```python
import numpy as np

kernel_name = "dist_sparse_attn_blocksparse_htp_b2_sq128_skv128_hq4_dh64"

def setup_inputs():
    x = np.random.randn(2, 128, 512).astype(np.float32)
    Wq = np.random.randn(512, 1024).astype(np.float32) * 0.02
    K_ext = np.random.randn(2, 128, 16, 64).astype(np.float32)
    V_ext = np.random.randn(2, 128, 16, 64).astype(np.float32)
    Wo = np.random.randn(1024, 512).astype(np.float32) * 0.02
    return {"x": x, "Wq": Wq, "K_ext": K_ext, "V_ext": V_ext, "Wo": Wo}

def reference(x, Wq, K_ext, V_ext, Wo):
    B, Sq, Skv, Hq, Dh = 2, 128, 128, 16, 64
    Q = (x @ Wq).reshape(B, Sq, Hq, Dh)
    qb = (np.arange(Sq) // 64)[:, None]
    kb = (np.arange(Skv) // 64)[None, :]
    mask = (qb == kb) | (kb == 0) | ((qb + kb) % 3 == 0)
    scores = np.einsum('bihd,bjhd->bhij', Q, K_ext).astype(np.float32) * 0.125
    scores = np.where(mask[None, None, :, :], scores, -1e9)
    scores_max = scores.max(axis=-1, keepdims=True)
    w = np.exp(scores - scores_max)
    row_keep = mask.any(axis=1)
    w_sum = np.where(row_keep[None, None, :, None], w.sum(axis=-1, keepdims=True), 1.0)
    w = w / w_sum
    w = np.where(row_keep[None, None, :, None], w, 0.0)
    ctx = np.einsum('bhij,bjhd->bihd', w, V_ext).reshape(B, Sq, Hq * Dh)
    return ctx @ Wo
```

```python
import math

import jax
import jax.numpy as jnp
from jax import lax
from jax.experimental import pallas as pl
from jax.experimental.pallas import tpu as pltpu

BF = jnp.bfloat16
F32 = jnp.float32
MESH = pl.DeviceIdType.MESH

C_EXP = 0.125 * math.log2(math.e)
MASK = -8e9
NP = 4
RP = 64 // NP
G = 16
WQ_SPLIT = ((0, 256), (256, 384), (384, 512))


def _body(x_hbm, wq_hbm, k_hbm, v_hbm, wo_hbm, o_ref,
          xs, wq, kb, vb, wo, qacc, acc, sb, rb, lsem, ssem, rsem1, rsem2, rsem3):
    def wqcp(i):
        a, b = WQ_SPLIT[i]
        sl = pl.ds(a, b - a)
        return pltpu.make_async_copy(wq_hbm.at[sl], wq.at[sl], lsem.at[12 + i])

    wqcp(0).start()
    p = lax.axis_index("i")
    cx = p >> 1
    cy = (p ^ cx) & 1
    diff = cx ^ cy
    part = (p ^ 1, 3 - p)
    rows = (cy * 128, cx * 128 + 64, (1 - cy) * 128, (1 - cx) * 128 + 64)
    hrow = pl.multiple_of(p * 256, 256)

    def xcp(r):
        return pltpu.make_async_copy(
            x_hbm.at[pl.ds(pl.multiple_of(rows[r], 64), 64)],
            xs.at[pl.ds(64 * r, 64)], lsem.at[r])

    def kcp(s):
        b = cy if s == 0 else 1 - cy
        return pltpu.make_async_copy(k_hbm.at[b, pl.ds(hrow, 256)], kb.at[s], lsem.at[4 + s])

    def vcp(s):
        b = cy if s == 0 else 1 - cy
        return pltpu.make_async_copy(v_hbm.at[b, pl.ds(hrow, 256)], vb.at[s], lsem.at[6 + s])

    def wocp(j):
        return pltpu.make_async_copy(wo_hbm.at[:, pl.ds(128 * j, 128)], wo.at[j], lsem.at[8 + j])

    def when(c, f):
        pl.when(c)(f)

    xcp(0).start()
    xcp(1).start()
    for i in range(1, len(WQ_SPLIT)):
        wqcp(i).start()
    kcp(0).start()
    when(diff == 1, lambda: kcp(1).start())
    vcp(0).start()
    when(diff == 1, lambda: vcp(1).start())
    wocp(0).start()
    wocp(1).start()
    xcp(2).start()
    xcp(3).start()
    wocp(2).start()
    when(diff == 0, lambda: kcp(1).start())
    wocp(3).start()
    when(diff == 0, lambda: vcp(1).start())
    bs = pltpu.get_barrier_semaphore()
    for n in part:
        pl.semaphore_signal(bs, inc=1, device_id=(n,), device_id_type=MESH)

    lane = lax.broadcasted_iota(jnp.int32, (64, 128), 1)
    lo = lane < 64
    z = jnp.zeros((64, 128), F32)

    def dot(a, b):
        return jnp.dot(a, b, preferred_element_type=F32)

    def scores(q, slot, masked):
        out = []
        for h in range(4):
            pr = h // 2
            kh = kb[slot, 64 * h:64 * h + 64, :]
            w = jnp.concatenate([kh, z] if h % 2 == 0 else [z, kh], 0)
            s = dot(q[:, 128 * pr:128 * pr + 128], w)
            if masked:
                s = jnp.where(lo, s, MASK)
            m = jnp.max(s, axis=1, keepdims=True)
            out.append(jnp.exp2((s - m) * C_EXP))
        return out

    def pv(ps, slot):
        ctxs = []
        for pr in range(2):
            w = vb[slot, 128 * pr:128 * pr + 128, :]
            p0, p1 = ps[2 * pr], ps[2 * pr + 1]
            lhs = jnp.concatenate(
                [t[g * G:(g + 1) * G] for g in range(64 // G) for t in (p0, p1)], 0)
            tt = lax.dot_general(lhs, w, (((1,), (1,)), ((), ())),
                                 preferred_element_type=F32)
            t = [jnp.concatenate([tt[(2 * g + i) * G:(2 * g + i + 1) * G]
                                  for g in range(64 // G)], 0) for i in range(2)]
            sm = [jnp.sum(pp, axis=1, keepdims=True) for pp in (p0, p1)]
            den = jnp.where(lo, sm[0], sm[1])
            r = pl.reciprocal(den, approx=True)
            r = r * (2.0 - den * r)
            ctxs.append(jnp.where(lo, t[0], t[1]) * r)
        return jnp.concatenate(ctxs, 1)

    def rcopy(step, half, j, n, sem):
        tgt = part[half] if step != 1 else part[1 - half]
        rs = pl.ds(n * RP, RP)
        return pltpu.make_async_remote_copy(
            src_ref=sb.at[step, half, j, rs], dst_ref=rb.at[step, half, j, rs],
            send_sem=ssem.at[step, half], recv_sem=sem.at[half, j, n],
            device_id=(tgt,), device_id_type=MESH)

    def oproj(ctx, j):
        w = wo[j]
        return [dot(ctx[half], w) for half in range(2)]

    def send1(o, j):
        for n in range(NP):
            for half in range(2):
                rs = slice(n * RP, (n + 1) * RP)
                sb[0, half, j, rs] = o[half][rs].astype(BF)
                rcopy(0, half, j, n, rsem1).start()

    nq = len(WQ_SPLIT)
    q0 = [None, None]
    for i, (a, b) in enumerate(WQ_SPLIT):
        wqcp(i).wait()
        if i == 0:
            xcp(0).wait()
            xcp(1).wait()
        if b - a > 128:
            xx = xs[0:128, a:b]
            tt = jnp.concatenate([dot(xx, wq[a:b, 0:128]), dot(xx, wq[a:b, 128:256])], 1)
        else:
            w = wq[a:b, :]
        for half in range(2):
            if b - a > 128:
                t = tt[64 * half:64 * half + 64]
            else:
                t = dot(xs[64 * half:64 * half + 64, a:b], w)
            if i > 0:
                t = t + qacc[half]
            if i < nq - 1:
                qacc[half] = t
            else:
                q0[half] = t
    kcp(0).wait()
    when(diff == 1, lambda: kcp(1).wait())
    pa = scores(q0[0], 0, True)
    pb = scores(q0[1], diff, False)
    vcp(0).wait()
    when(diff == 1, lambda: vcp(1).wait())
    wocp(0).wait()
    pl.semaphore_wait(bs, 2)
    ctx0 = [pv(pa, 0), pv(pb, diff)]
    send1(oproj(ctx0, 0), 0)
    wocp(1).wait()
    send1(oproj(ctx0, 1), 1)

    xcp(2).wait()
    xcp(3).wait()
    q = dot(xs[128:256, :], wq[...])
    wocp(2).wait()
    when(diff == 0, lambda: kcp(1).wait())
    o = oproj(ctx0, 2)
    pa = scores(q[0:64], 1, True)
    pb = scores(q[64:128], 1 - diff, False)
    send1(o, 2)
    wocp(3).wait()
    when(diff == 0, lambda: vcp(1).wait())
    o = oproj(ctx0, 3)
    ctx1 = jnp.concatenate([pv(pa, 1), pv(pb, 1 - diff)], 0)
    oo = [dot(ctx1, wo[j]) for j in range(4)]
    send1(o, 3)
    for j in range(4):
        acc[0, j] = oo[j][0:64]
        acc[1, j] = oo[j][64:128]

    for j in range(4):
        for n in range(NP):
            rs = slice(n * RP, (n + 1) * RP)
            for half in range(2):
                rcopy(0, half, j, n, rsem1).wait_recv()
                a = acc[half, j, rs] + rb[0, half, j, rs].astype(F32)
                sb[1, half, j, rs] = a.astype(BF)
                rcopy(1, half, j, n, rsem2).start()
                acc[half, j, rs] = a

    for j in range(4):
        for n in range(NP):
            rs = slice(n * RP, (n + 1) * RP)
            for half in range(2):
                rcopy(1, half, j, n, rsem2).wait_recv()
                t = acc[half, j, rs] + rb[1, half, j, rs].astype(F32)
                sb[2, half, j, rs] = t.astype(BF)
                rcopy(2, half, j, n, rsem3).start()
                r0 = pl.multiple_of(rows[2 + half] + n * RP, RP)
                o_ref[pl.ds(r0, RP), 128 * j:128 * j + 128] = t
    for j in range(4):
        for n in range(NP):
            rs = slice(n * RP, (n + 1) * RP)
            for half in range(2):
                rcopy(2, half, j, n, rsem3).wait_recv()
                r0 = pl.multiple_of(rows[half] + n * RP, RP)
                o_ref[pl.ds(r0, RP), 128 * j:128 * j + 128] = rb[2, half, j, rs].astype(F32)
    for step in range(3):
        for half in range(2):
            pltpu.make_async_copy(sb.at[step, half], sb.at[step, half], ssem.at[step, half]).wait()


def pallas_dist_sparse_attn_blocksparse_htp_b2_sq128_skv128_hq4_dh64_kernel(
    x: jax.Array,
    Wq: jax.Array,
    K_ext: jax.Array,
    V_ext: jax.Array,
    Wo: jax.Array,
):
    kt = jnp.transpose(K_ext, (0, 2, 3, 1)).reshape(2, 1024, 128)
    vt = jnp.transpose(V_ext, (0, 2, 3, 1)).reshape(2, 1024, 128)
    x2 = x.reshape(256, 512)
    any_ = pl.BlockSpec(memory_space=pl.ANY)
    out = pl.pallas_call(
        _body,
        out_shape=jax.ShapeDtypeStruct((256, 512), F32),
        in_specs=[any_] * 5,
        out_specs=pl.BlockSpec(memory_space=pltpu.VMEM),
        scratch_shapes=[
            pltpu.VMEM((256, 512), F32),
            pltpu.VMEM((512, 256), F32),
            pltpu.VMEM((2, 256, 128), F32),
            pltpu.VMEM((2, 256, 128), F32),
            pltpu.VMEM((4, 256, 128), F32),
            pltpu.VMEM((2, 64, 256), F32),
            pltpu.VMEM((2, 4, 64, 128), F32),
            pltpu.VMEM((3, 2, 4, 64, 128), BF),
            pltpu.VMEM((3, 2, 4, 64, 128), BF),
            pltpu.SemaphoreType.DMA((15,)),
            pltpu.SemaphoreType.DMA((3, 2)),
            pltpu.SemaphoreType.DMA((2, 4, NP)),
            pltpu.SemaphoreType.DMA((2, 4, NP)),
            pltpu.SemaphoreType.DMA((2, 4, NP)),
        ],
        compiler_params=pltpu.CompilerParams(
            collective_id=0,
            disable_semaphore_checks=True,
            disable_bounds_checks=True,
        ),
    )(x2, Wq, kt, vt, Wo)
    return out.reshape(2, 128, 512)
```

```python
import functools
import math

import jax
import jax.numpy as jnp
from jax import lax
from jax.experimental import pallas as pl
from jax.experimental.pallas import tpu as pltpu

BF = jnp.bfloat16
F32 = jnp.float32
MESH = pl.DeviceIdType.MESH

C_EXP = 0.125 * math.log2(math.e)
MASK = -8e9
RP = 8
NP = 64 // RP
G = 16
XS = 32
WQ_SPLIT = ((0, 256), (256, 384), (384, 512))


def _program(p, x_hbm, wq_hbm, k_hbm, v_hbm, wo_hbm, o_ref,
             xs, wq, kb, vb, wo, qacc, acc, sb, rb, sbx, rbx,
             lsem, ssem, rsem1, rsem2, rsem3, xssem, xrsem):
    cx = p >> 1
    cy = (p ^ cx) & 1
    part = (p ^ 1, 3 - p)
    batch = (cy, cx, 1 - cy, 1 - cx)
    rows = tuple(batch[c] * 128 + 64 * (c % 2) for c in range(4))
    role = "AMZM"[p]
    f = 1 if p == 3 else 0
    g = 1 - f
    xsend = {"A": (0, 1), "M": (g,), "Z": ()}[role]
    xrecv = {"A": (), "M": (f,), "Z": (0, 1)}[role]

    def load_wq(i, sem):
        a, b = WQ_SPLIT[i]
        sl = pl.ds(a, b - a)
        return pltpu.make_async_copy(wq_hbm.at[sl], wq.at[sl], sem)

    def load_x(c, sem):
        r0 = XS if c - 2 in xrecv else 0
        return pltpu.make_async_copy(x_hbm.at[pl.ds(rows[c] + r0, 64 - r0)],
                                     xs.at[pl.ds(64 * c + r0, 64 - r0)], sem)

    def load_kv(src, dst, i, sem):
        b = batch[f] if i == 0 else 1 - batch[f]
        return pltpu.make_async_copy(src.at[b, pl.ds(p * 256, 256)], dst.at[b], sem)

    def load_wo(j, sem):
        sl = pl.ds(128 * j, 128)
        return pltpu.make_async_copy(wo_hbm.at[:, sl], wo.at[:, sl], sem)

    makers = {"q": load_wq, "x": load_x, "w": load_wo,
              "k": functools.partial(load_kv, k_hbm, kb),
              "v": functools.partial(load_kv, v_hbm, vb)}
    order = {
        "A": "q0 x0 x1 q1 q2 k0 v0 w0 w1 x2 x3 w2 k1 w3 v1",
        "M": f"q0 x0 x1 q1 q2 k0 k1 v0 v1 w0 w1 x{2 + g} x{2 + f} w2 w3",
        "Z": "q0 x0 x1 q1 q2 k0 v0 w0 w1 w2 x2 x3 w3 k1 v1",
    }[role].split()
    barrier = pltpu.get_barrier_semaphore()
    loads = {}
    for ix, nm in enumerate(order):
        loads[nm] = makers[nm[0]](int(nm[1]), lsem.at[ix])
        loads[nm].start()
        if ix == 0:
            for n in part:
                pl.semaphore_signal(barrier, inc=1, device_id=(n,), device_id_type=MESH)

    def wait(names):
        for nm in names.split():
            loads.pop(nm).wait()

    rsems = (rsem1, rsem2, rsem3)

    def rcopy(step, half, j, n):
        tgt = part[half] if step != 1 else part[1 - half]
        rs = pl.ds(n * RP, RP)
        return pltpu.make_async_remote_copy(
            src_ref=sb.at[step, half, j, rs], dst_ref=rb.at[step, half, j, rs],
            send_sem=ssem.at[step, half], recv_sem=rsems[step].at[half, j, n],
            device_id=(tgt,), device_id_type=MESH)

    def xcopy(half):
        return pltpu.make_async_remote_copy(
            src_ref=sbx.at[half], dst_ref=rbx.at[half],
            send_sem=xssem.at[half], recv_sem=xrsem.at[half],
            device_id=(part[half],), device_id_type=MESH)

    def enter():
        pl.semaphore_wait(barrier, 2)
        for half in xsend:
            xcopy(half).start()

    lo = lax.broadcasted_iota(jnp.int32, (64, 128), 1) < 64
    zero = jnp.zeros((64, 128), F32)
    q, prob, ctx, out = {}, {}, {}, {}

    def dot(a, b):
        return jnp.dot(a, b, preferred_element_type=F32)

    def scores(c):
        prob[c] = []
        for h in range(4):
            pr = h // 2
            kh = kb[batch[c], 64 * h:64 * h + 64, :]
            w = jnp.concatenate([kh, zero] if h % 2 == 0 else [zero, kh], 0)
            s = dot(q[c][:, 128 * pr:128 * pr + 128], w)
            if c % 2 == 0:
                s = jnp.where(lo, s, MASK)
            m = jnp.max(s, axis=1, keepdims=True)
            prob[c].append(jnp.exp2((s - m) * C_EXP))

    def pv(c):
        cs = []
        for pr in range(2):
            w = vb[batch[c], 128 * pr:128 * pr + 128, :]
            pp = prob[c][2 * pr:2 * pr + 2]
            lhs = jnp.concatenate(
                [t[u * G:(u + 1) * G] for u in range(64 // G) for t in pp], 0)
            tt = lax.dot_general(lhs, w, (((1,), (1,)), ((), ())),
                                 preferred_element_type=F32)
            t = [jnp.concatenate([tt[(2 * u + i) * G:(2 * u + i + 1) * G]
                                  for u in range(64 // G)], 0) for i in range(2)]
            sm = [jnp.sum(a, axis=1, keepdims=True) for a in pp]
            den = jnp.where(lo, sm[0], sm[1])
            r = pl.reciprocal(den, approx=True)
            r = r * (2.0 - den * r)
            cs.append(jnp.where(lo, t[0], t[1]) * r)
        ctx[c] = jnp.concatenate(cs, 1)

    def oproj(c, j):
        out[c, j] = dot(ctx[c], wo[:, 128 * j:128 * j + 128])

    def oproj_kept(j):
        o = dot(jnp.concatenate([ctx[2], ctx[3]], 0), wo[:, 128 * j:128 * j + 128])
        out[2, j], out[3, j] = o[0:64], o[64:128]

    def oproj_sent(j):
        oproj(f, j)
        oproj(g, j)

    def q_kept():
        xx = []
        for c in (2, 3):
            if c - 2 in xrecv:
                xx += [jnp.concatenate([rbx[c - 2, u, j].astype(F32) for j in range(4)], 1)
                       for u in range(XS // 16)]
                xx.append(xs[64 * c + XS:64 * c + 64, :])
            else:
                xx.append(xs[64 * c:64 * c + 64, :])
        t = dot(jnp.concatenate(xx, 0), wq[...])
        q[2], q[3] = t[0:64], t[64:128]

    def wait_x():
        for half in xrecv:
            xcopy(half).wait_recv()

    def step1(j):
        for n in range(NP):
            rs = slice(n * RP, (n + 1) * RP)
            for half in (f, g):
                sb[0, half, j, rs] = out[half, j][rs].astype(BF)
                rcopy(0, half, j, n).start()

    def keep(j, r0=0):
        for c in (2, 3):
            acc[c - 2, j, r0:64] = out[c, j][r0:64]

    done = set()

    def step2(j, n, direct=False):
        rs = slice(n * RP, (n + 1) * RP)
        for half in range(2):
            if direct:
                own = out[2 + half, j][rs]
            else:
                rcopy(0, half, j, n).wait_recv()
                own = acc[half, j, rs]
            a = own + rb[0, half, j, rs].astype(F32)
            sb[1, half, j, rs] = a.astype(BF)
            rcopy(1, half, j, n).start()
            acc[half, j, rs] = a
        done.add((j, n))

    for i, (a, b) in enumerate(WQ_SPLIT):
        if role == "M" and i == 1:
            enter()
        wait("q0 x0 x1" if i == 0 else f"q{i}")
        if i == 0:
            for half in xsend:
                for u in range(XS // 16):
                    r0 = 64 * half + 16 * u
                    for j in range(4):
                        sbx[half, u, j] = xs[r0:r0 + 16, 128 * j:128 * j + 128].astype(BF)
            xx = xs[0:128, a:b]
            tt = jnp.concatenate([dot(xx, wq[a:b, 0:128]), dot(xx, wq[a:b, 128:256])], 1)
        else:
            w = wq[a:b, :]
        for half in (f, g):
            if i == 0:
                t = tt[64 * half:64 * half + 64]
            else:
                t = dot(xs[64 * half:64 * half + 64, a:b], w) + qacc[half]
            if i < len(WQ_SPLIT) - 1:
                qacc[half] = t
            else:
                q[half] = t

    if role == "A":
        wait("k0")
        enter()
        scores(f), scores(g)
        wait("v0 w0")
        pv(f), pv(g), oproj_sent(0), step1(0)
        wait("w1")
        oproj_sent(1), step1(1)
        wait("x2 x3")
        q_kept()
        wait("w2 k1")
        oproj_sent(2), scores(2), scores(3), step1(2)
        wait("w3 v1")
        oproj_sent(3), pv(2), pv(3)
        for j in range(4):
            oproj_kept(j)
        step1(3)
        for j in range(4):
            keep(j)
    elif role == "M":
        wait("k0 k1")
        scores(f), scores(g)
        wait("v0 v1")
        pv(f), pv(g)
        wait("w0")
        oproj_sent(0), step1(0)
        wait("w1")
        oproj_sent(1), step1(1)
        wait(f"x{2 + g} x{2 + f}")
        wait_x()
        q_kept()
        wait("w2")
        oproj_sent(2), scores(2), scores(3), step1(2)
        wait("w3")
        oproj_sent(3), pv(2), pv(3)
        for j in range(4):
            oproj_kept(j)
        step1(3)
        for j in range(4):
            keep(j)
    else:
        wait("k0")
        scores(f), scores(g)
        wait("v0 w0")
        enter()
        pv(f), pv(g), oproj_sent(0), step1(0)
        wait("w1")
        oproj_sent(1), step1(1)
        wait("w2")
        oproj_sent(2), step1(2)
        wait("x2 x3")
        wait_x()
        q_kept()
        wait("w3 k1")
        oproj_sent(3), scores(2), scores(3), step1(3)
        wait("v1")
        for n0 in (0, 2):
            for half in range(2):
                for n in (n0, n0 + 1):
                    rcopy(0, half, 0, n).wait_recv()
        pv(2), pv(3)
        oproj(2, 0), oproj(3, 0), oproj(2, 1), oproj(3, 1)
        for n in range(4):
            step2(0, n, direct=True)
        keep(0, 4 * RP), keep(1)
        for j, n in [(0, n) for n in range(4, 8)] + [(1, n) for n in range(4)]:
            step2(j, n)
        oproj_kept(2), oproj_kept(3), keep(2), keep(3)
    assert not loads

    pieces = [(j, n) for j in range(4) for n in range(NP)]
    for j, n in pieces:
        if (j, n) not in done:
            step2(j, n)

    for j, n in pieces:
        rs = slice(n * RP, (n + 1) * RP)
        for half in range(2):
            rcopy(1, half, j, n).wait_recv()
            t = acc[half, j, rs] + rb[1, half, j, rs].astype(F32)
            sb[2, half, j, rs] = t.astype(BF)
            rcopy(2, half, j, n).start()
            o_ref[pl.ds(rows[2 + half] + n * RP, RP), 128 * j:128 * j + 128] = t

    for j, n in pieces:
        if (j, n) == pieces[-2]:
            for half in xsend:
                xcopy(half).wait_send()
            for step in range(3):
                for half in range(2):
                    pltpu.make_async_copy(sb.at[step, half], sb.at[step, half],
                                          ssem.at[step, half]).wait()
        rs = slice(n * RP, (n + 1) * RP)
        for half in range(2):
            rcopy(2, half, j, n).wait_recv()
            o_ref[pl.ds(rows[half] + n * RP, RP), 128 * j:128 * j + 128] = (
                rb[2, half, j, rs].astype(F32))


def _body(*refs):
    p = lax.axis_index("i")
    for ps in (2, 1, 3, 0):
        pl.when(p == ps)(functools.partial(_program, ps, *refs))


def pallas_dist_sparse_attn_blocksparse_htp_b2_sq128_skv128_hq4_dh64_kernel(
    x: jax.Array,
    Wq: jax.Array,
    K_ext: jax.Array,
    V_ext: jax.Array,
    Wo: jax.Array,
):
    kt = jnp.transpose(K_ext, (0, 2, 3, 1)).reshape(2, 1024, 128)
    vt = jnp.transpose(V_ext, (0, 2, 3, 1)).reshape(2, 1024, 128)
    x2 = x.reshape(256, 512)
    any_ = pl.BlockSpec(memory_space=pl.ANY)
    out = pl.pallas_call(
        _body,
        out_shape=jax.ShapeDtypeStruct((256, 512), F32),
        in_specs=[any_] * 5,
        out_specs=pl.BlockSpec(memory_space=pltpu.VMEM),
        scratch_shapes=[
            pltpu.VMEM((256, 512), F32),
            pltpu.VMEM((512, 256), F32),
            pltpu.VMEM((2, 256, 128), F32),
            pltpu.VMEM((2, 256, 128), F32),
            pltpu.VMEM((256, 512), F32),
            pltpu.VMEM((2, 64, 256), F32),
            pltpu.VMEM((2, 4, 64, 128), F32),
            pltpu.VMEM((3, 2, 4, 64, 128), BF),
            pltpu.VMEM((3, 2, 4, 64, 128), BF),
            pltpu.VMEM((2, XS // 16, 4, 16, 128), BF),
            pltpu.VMEM((2, XS // 16, 4, 16, 128), BF),
            pltpu.SemaphoreType.DMA((15,)),
            pltpu.SemaphoreType.DMA((3, 2)),
            pltpu.SemaphoreType.DMA((2, 4, NP)),
            pltpu.SemaphoreType.DMA((2, 4, NP)),
            pltpu.SemaphoreType.DMA((2, 4, NP)),
            pltpu.SemaphoreType.DMA((2,)),
            pltpu.SemaphoreType.DMA((2,)),
        ],
        compiler_params=pltpu.CompilerParams(
            collective_id=0,
            disable_semaphore_checks=True,
            disable_bounds_checks=True,
        ),
    )(x2, Wq, kt, vt, Wo)
    return out.reshape(2, 128, 512)
```

```python
import functools
import math

import jax
import jax.numpy as jnp
from jax import lax
from jax.experimental import pallas as pl
from jax.experimental.pallas import tpu as pltpu

BF = jnp.bfloat16
F32 = jnp.float32
MESH = pl.DeviceIdType.MESH

C_EXP = 0.125 * math.log2(math.e)
MASK = -8e9
RP = 8
NP = 64 // RP
G = 16
WQ_SPLIT = ((0, 256), (256, 384), (384, 512))
X_FWD = {"A": 48, "M": 32}
DETOUR = ((0, 2), (0, 3))
N_DIRECT = 2


def _program(p, x_hbm, wq_hbm, k_hbm, v_hbm, wo_hbm, o_ref,
             xs, wq, kb, vb, wo, qacc, acc, sb, rb, sbx, rbx, rbd,
             lsem, ssem, rsem1, rsem2, rsem3, xssem, xrsem, dsem):
    cx = p >> 1
    cy = (p ^ cx) & 1
    part = (p ^ 1, 3 - p)
    batch = (cy, cx, 1 - cy, 1 - cx)
    rows = tuple(batch[c] * 128 + 64 * (c % 2) for c in range(4))
    role = "AMZM"[p]
    f = 1 if p == 3 else 0
    g = 1 - f
    xsend = {"A": (0, 1), "M": (g,), "Z": ()}[role]
    xrecv = {"A": (), "M": (f,), "Z": (0, 1)}[role]
    n_xsend = X_FWD.get(role, 0)
    n_xrecv = {"A": 0, "M": X_FWD["A"], "Z": X_FWD["M"]}[role]
    pieces = [(j, n) for j in range(4) for n in range(NP)]
    z_order = [s for s in pieces[NP:] + pieces[:NP] if s not in DETOUR] + list(DETOUR)

    def load_wq(i, sem):
        a, b = WQ_SPLIT[i]
        sl = pl.ds(a, b - a)
        return pltpu.make_async_copy(wq_hbm.at[sl], wq.at[sl], sem)

    def load_x(c, sem):
        r0 = n_xrecv if c - 2 in xrecv else 0
        return pltpu.make_async_copy(x_hbm.at[pl.ds(rows[c] + r0, 64 - r0)],
                                     xs.at[pl.ds(64 * c + r0, 64 - r0)], sem)

    def load_kv(src, dst, i, sem):
        b = batch[f] if i == 0 else 1 - batch[f]
        return pltpu.make_async_copy(src.at[b, pl.ds(p * 256, 256)], dst.at[b], sem)

    def load_wo(j, sem):
        sl = pl.ds(128 * j, 128)
        return pltpu.make_async_copy(wo_hbm.at[:, sl], wo.at[:, sl], sem)

    makers = {"q": load_wq, "x": load_x, "w": load_wo,
              "k": functools.partial(load_kv, k_hbm, kb),
              "v": functools.partial(load_kv, v_hbm, vb)}
    order = {
        "A": "q0 x0 x1 q1 q2 k0 v0 w0 w1 x2 x3 w2 k1 w3 v1",
        "M": f"q0 x0 x1 q1 q2 k0 k1 v0 v1 w0 w1 w2 x{2 + g} x{2 + f} w3",
        "Z": "q0 x0 x1 q1 q2 k0 v0 w1 w2 w3 x2 x3 w0 k1 v1",
    }[role].split()
    barrier = pltpu.get_barrier_semaphore()
    loads = {}
    for ix, nm in enumerate(order):
        loads[nm] = makers[nm[0]](int(nm[1]), lsem.at[ix])
        loads[nm].start()
        if ix == 0:
            for n in part:
                pl.semaphore_signal(barrier, inc=1, device_id=(n,), device_id_type=MESH)

    def wait(names):
        for nm in names.split():
            loads.pop(nm).wait()

    rsems = (rsem1, rsem2, rsem3)

    def rcopy(step, half, j, n):
        tgt = part[half] if step != 1 else part[1 - half]
        rs = pl.ds(n * RP, RP)
        return pltpu.make_async_remote_copy(
            src_ref=sb.at[step, half, j, rs], dst_ref=rb.at[step, half, j, rs],
            send_sem=ssem.at[step, half], recv_sem=rsems[step].at[half, j, n],
            device_id=(tgt,), device_id_type=MESH)

    def dcopy(half, j, n):
        i = DETOUR.index((j, n))
        return pltpu.make_async_remote_copy(
            src_ref=sb.at[0, half, j, pl.ds(n * RP, RP)], dst_ref=rbd.at[half, pl.ds(i * RP, RP)],
            send_sem=ssem.at[0, half], recv_sem=dsem.at[half, i],
            device_id=(part[1 - half],), device_id_type=MESH)

    def xcopy(half, n):
        return pltpu.make_async_remote_copy(
            src_ref=sbx.at[half, pl.ds(0, n // 16)], dst_ref=rbx.at[half, pl.ds(0, n // 16)],
            send_sem=xssem.at[half], recv_sem=xrsem.at[half],
            device_id=(part[half],), device_id_type=MESH)

    def enter():
        pl.semaphore_wait(barrier, 2)
        for half in xsend:
            xcopy(half, n_xsend).start()

    lo = lax.broadcasted_iota(jnp.int32, (64, 128), 1) < 64
    zero = jnp.zeros((64, 128), F32)
    q, prob, ctx, out = {}, {}, {}, {}

    def dot(a, b):
        return jnp.dot(a, b, preferred_element_type=F32)

    def scores(c):
        prob[c] = []
        for h in range(4):
            pr = h // 2
            kh = kb[batch[c], 64 * h:64 * h + 64, :]
            w = jnp.concatenate([kh, zero] if h % 2 == 0 else [zero, kh], 0)
            s = dot(q[c][:, 128 * pr:128 * pr + 128], w)
            if c % 2 == 0:
                s = jnp.where(lo, s, MASK)
            m = jnp.max(s, axis=1, keepdims=True)
            prob[c].append(jnp.exp2((s - m) * C_EXP))

    def pv(c):
        cs = []
        for pr in range(2):
            w = vb[batch[c], 128 * pr:128 * pr + 128, :]
            pp = prob[c][2 * pr:2 * pr + 2]
            lhs = jnp.concatenate(
                [t[u * G:(u + 1) * G] for u in range(64 // G) for t in pp], 0)
            tt = lax.dot_general(lhs, w, (((1,), (1,)), ((), ())),
                                 preferred_element_type=F32)
            t = [jnp.concatenate([tt[(2 * u + i) * G:(2 * u + i + 1) * G]
                                  for u in range(64 // G)], 0) for i in range(2)]
            sm = [jnp.sum(a, axis=1, keepdims=True) for a in pp]
            den = jnp.where(lo, sm[0], sm[1])
            r = pl.reciprocal(den, approx=True)
            r = r * (2.0 - den * r)
            cs.append(jnp.where(lo, t[0], t[1]) * r)
        ctx[c] = jnp.concatenate(cs, 1)

    def oproj(c, j):
        out[c, j] = dot(ctx[c], wo[:, 128 * j:128 * j + 128])

    def oproj_kept(j):
        o = dot(jnp.concatenate([ctx[2], ctx[3]], 0), wo[:, 128 * j:128 * j + 128])
        out[2, j], out[3, j] = o[0:64], o[64:128]

    def oproj_sent(j):
        oproj(f, j)
        oproj(g, j)

    def q_kept():
        xx = []
        for c in (2, 3):
            if c - 2 in xrecv:
                xx += [jnp.concatenate([rbx[c - 2, u, j].astype(F32) for j in range(4)], 1)
                       for u in range(n_xrecv // 16)]
                xx.append(xs[64 * c + n_xrecv:64 * c + 64, :])
            else:
                xx.append(xs[64 * c:64 * c + 64, :])
        t = dot(jnp.concatenate(xx, 0), wq[...])
        q[2], q[3] = t[0:64], t[64:128]

    def wait_x():
        for half in xrecv:
            xcopy(half, n_xrecv).wait_recv()

    def keep(j, r0=0):
        for c in (2, 3):
            acc[c - 2, j, r0:64] = out[c, j][r0:64]

    def store(c, j, n, t):
        o_ref[pl.ds(rows[c] + n * RP, RP), 128 * j:128 * j + 128] = t

    def step1(j):
        for n in range(NP):
            rs = slice(n * RP, (n + 1) * RP)
            detour = (j, n) in DETOUR
            for half in (f, g):
                if detour and role == "Z":
                    continue
                sb[0, half, j, rs] = out[half, j][rs].astype(BF)
                if detour and role == "M" and half == f:
                    dcopy(half, j, n).start()
                else:
                    rcopy(0, half, j, n).start()

    def step1_detour():
        for i, (j, n) in enumerate(DETOUR):
            rs = slice(n * RP, (n + 1) * RP)
            for half in range(2):
                a = out[half, j][rs] + rbd[half, i * RP:(i + 1) * RP].astype(F32)
                sb[0, half, j, rs] = a.astype(BF)
                rcopy(0, half, j, n).start()

    done2, done3 = set(), set()

    def step2(half, j, n, direct=False):
        rs = slice(n * RP, (n + 1) * RP)
        detour = (j, n) in DETOUR
        done2.add((half, j, n))
        if detour and role == "A":
            sb[1, half, j, rs] = acc[half, j, rs].astype(BF)
            rcopy(1, half, j, n).start()
        elif detour and role == "M" and half == g:
            rcopy(1, half, j, n).wait_recv()
            rcopy(0, half, j, n).wait_recv()
            t = (acc[half, j, rs] + rb[1, half, j, rs].astype(F32)
                 + rb[0, half, j, rs].astype(F32))
            for step in (1, 2):
                sb[step, half, j, rs] = t.astype(BF)
                rcopy(step, half, j, n).start()
            store(2 + half, j, n, t)
            done3.add((half, j, n))
        else:
            if direct:
                own = out[2 + half, j][rs]
            else:
                rcopy(0, half, j, n).wait_recv()
                own = acc[half, j, rs]
            a = own + rb[0, half, j, rs].astype(F32)
            sb[1, half, j, rs] = a.astype(BF)
            rcopy(1, half, j, n).start()
            acc[half, j, rs] = a

    def step3(half, j, n):
        rs = slice(n * RP, (n + 1) * RP)
        rcopy(1, half, j, n).wait_recv()
        t = rb[1, half, j, rs].astype(F32)
        if not ((j, n) in DETOUR and role == "A"):
            t = acc[half, j, rs] + t
        sb[2, half, j, rs] = t.astype(BF)
        rcopy(2, half, j, n).start()
        store(2 + half, j, n, t)

    for i, (a, b) in enumerate(WQ_SPLIT):
        if role == "M" and i == 1:
            enter()
        wait("q0 x0 x1" if i == 0 else f"q{i}")
        if i == 0:
            for half in xsend:
                for u in range(n_xsend // 16):
                    r0 = 64 * half + 16 * u
                    for j in range(4):
                        sbx[half, u, j] = xs[r0:r0 + 16, 128 * j:128 * j + 128].astype(BF)
            xx = xs[0:128, a:b]
            tt = jnp.concatenate([dot(xx, wq[a:b, 0:128]), dot(xx, wq[a:b, 128:256])], 1)
        else:
            w = wq[a:b, :]
        for half in (f, g):
            if i == 0:
                t = tt[64 * half:64 * half + 64]
            else:
                t = dot(xs[64 * half:64 * half + 64, a:b], w) + qacc[half]
            if i < len(WQ_SPLIT) - 1:
                qacc[half] = t
            else:
                q[half] = t

    if role == "A":
        wait("k0")
        enter()
        scores(f), scores(g)
        wait("v0 w0")
        pv(f), pv(g), oproj_sent(0), step1(0)
        wait("w1")
        oproj_sent(1), step1(1)
        wait("x2 x3")
        q_kept()
        wait("w2 k1")
        oproj_sent(2), scores(2), scores(3), step1(2)
        wait("w3 v1")
        oproj_sent(3), pv(2), pv(3)
        for j in range(4):
            oproj_kept(j)
        step1(3)
        for j in range(4):
            keep(j)
    elif role == "M":
        wait("k0 k1")
        scores(f), scores(g)
        wait("v0 v1")
        pv(f), pv(g)
        for j in range(3):
            wait(f"w{j}")
            oproj_sent(j), step1(j)
        wait(f"x{2 + g} x{2 + f}")
        wait_x()
        q_kept()
        wait("w3")
        scores(2), scores(3), oproj_sent(3), pv(2), pv(3), step1(3)
        for c in (2, 3):
            for j in range(4):
                oproj(c, j)
        for j in range(4):
            keep(j)
    else:
        wait("k0")
        scores(f), scores(g)
        wait("v0 w1")
        enter()
        pv(f), pv(g), oproj_sent(1), step1(1)
        wait("w2")
        oproj_sent(2), step1(2)
        wait("w3 x2 x3")
        wait_x()
        oproj_sent(3), q_kept(), step1(3)
        wait("w0 k1")
        scores(2), scores(3), oproj_sent(0), step1(0)
        wait("v1")
        for half in range(2):
            for n in range(N_DIRECT):
                rcopy(0, half, 0, n).wait_recv()
            for j, n in DETOUR:
                dcopy(half, j, n).wait_recv()
        pv(2), pv(3), step1_detour()
        oproj(2, 0), oproj(3, 0), oproj(2, 1), oproj(3, 1)
        for n in range(N_DIRECT):
            for half in range(2):
                step2(half, 0, n, direct=True)
        keep(0, N_DIRECT * RP), keep(1)
        for j, n in pieces[N_DIRECT:NP + NP // 2]:
            for half in range(2):
                step2(half, j, n)
        oproj_kept(2), oproj_kept(3), keep(2), keep(3)
    assert not loads

    for t in range(len(pieces)):
        for half in range(2):
            j, n = (z_order if role == "M" and half == g else pieces)[t]
            if (half, j, n) not in done2:
                step2(half, j, n)

    for t in range(len(pieces)):
        for half in range(2):
            j, n = (z_order if role == "A" else pieces)[t]
            if (half, j, n) not in done3:
                step3(half, j, n)

    for t in range(len(pieces)):
        if t == len(pieces) - 2:
            for half in xsend:
                xcopy(half, n_xsend).wait_send()
            for step in range(3):
                for half in range(2):
                    pltpu.make_async_copy(sb.at[step, half], sb.at[step, half],
                                          ssem.at[step, half]).wait()
        for half in range(2):
            j, n = (z_order if role == "M" and half == f else pieces)[t]
            rcopy(2, half, j, n).wait_recv()
            store(half, j, n, rb[2, half, j, n * RP:(n + 1) * RP].astype(F32))


def _body(*refs):
    p = lax.axis_index("i")
    for ps in (2, 1, 3, 0):
        pl.when(p == ps)(functools.partial(_program, ps, *refs))


def pallas_dist_sparse_attn_blocksparse_htp_b2_sq128_skv128_hq4_dh64_kernel(
    x: jax.Array,
    Wq: jax.Array,
    K_ext: jax.Array,
    V_ext: jax.Array,
    Wo: jax.Array,
):
    kt = jnp.transpose(K_ext, (0, 2, 3, 1)).reshape(2, 1024, 128)
    vt = jnp.transpose(V_ext, (0, 2, 3, 1)).reshape(2, 1024, 128)
    x2 = x.reshape(256, 512)
    any_ = pl.BlockSpec(memory_space=pl.ANY)
    nx = max(X_FWD.values()) // 16
    out = pl.pallas_call(
        _body,
        out_shape=jax.ShapeDtypeStruct((256, 512), F32),
        in_specs=[any_] * 5,
        out_specs=pl.BlockSpec(memory_space=pltpu.VMEM),
        scratch_shapes=[
            pltpu.VMEM((256, 512), F32),
            pltpu.VMEM((512, 256), F32),
            pltpu.VMEM((2, 256, 128), F32),
            pltpu.VMEM((2, 256, 128), F32),
            pltpu.VMEM((256, 512), F32),
            pltpu.VMEM((2, 64, 256), F32),
            pltpu.VMEM((2, 4, 64, 128), F32),
            pltpu.VMEM((3, 2, 4, 64, 128), BF),
            pltpu.VMEM((3, 2, 4, 64, 128), BF),
            pltpu.VMEM((2, nx, 4, 16, 128), BF),
            pltpu.VMEM((2, nx, 4, 16, 128), BF),
            pltpu.VMEM((2, len(DETOUR) * RP, 128), BF),
            pltpu.SemaphoreType.DMA((15,)),
            pltpu.SemaphoreType.DMA((3, 2)),
            pltpu.SemaphoreType.DMA((2, 4, NP)),
            pltpu.SemaphoreType.DMA((2, 4, NP)),
            pltpu.SemaphoreType.DMA((2, 4, NP)),
            pltpu.SemaphoreType.DMA((2,)),
            pltpu.SemaphoreType.DMA((2,)),
            pltpu.SemaphoreType.DMA((2, len(DETOUR))),
        ],
        compiler_params=pltpu.CompilerParams(
            collective_id=0,
            disable_semaphore_checks=True,
            disable_bounds_checks=True,
        ),
    )(x2, Wq, kt, vt, Wo)
    return out.reshape(2, 128, 512)
```

```python
import functools
import math

import jax
import jax.numpy as jnp
from jax import lax
from jax.experimental import pallas as pl
from jax.experimental.pallas import tpu as pltpu

BF = jnp.bfloat16
F32 = jnp.float32
MESH = pl.DeviceIdType.MESH

C_EXP = 0.125 * math.log2(math.e)
MASK = -8e9
RP = 8
NP = 64 // RP
G = 16
WQ_SPLIT = ((0, 256), (256, 384), (384, 512))
X_FWD = {"A": 48, "M": 32}
DETOUR = ((0, 2), (0, 3))
N_DIRECT = 3


def _program(p, x_hbm, wq_hbm, k_hbm, v_hbm, wo_hbm, o_ref,
             xs, wq, kb, vb, wo, wo12, qacc, acc, sb, rb, sbx, rbx, rbd,
             lsem, ssem, rsem1, rsem2, rsem3, xssem, xrsem, dsem):
    cx = p >> 1
    cy = (p ^ cx) & 1
    part = (p ^ 1, 3 - p)
    batch = (cy, cx, 1 - cy, 1 - cx)
    rows = tuple(batch[c] * 128 + 64 * (c % 2) for c in range(4))
    role = "AMZM"[p]
    f = 1 if p == 3 else 0
    g = 1 - f
    xsend = {"A": (0, 1), "M": (g,), "Z": ()}[role]
    xrecv = {"A": (), "M": (f,), "Z": (0, 1)}[role]
    n_xsend = X_FWD.get(role, 0)
    n_xrecv = {"A": 0, "M": X_FWD["A"], "Z": X_FWD["M"]}[role]
    pieces = [(j, n) for j in range(4) for n in range(NP)]
    z_order = [(j, n) for j in (3, 1, 2, 0) for n in range(NP) if (j, n) not in DETOUR]
    z_order += list(DETOUR)

    def load_wq(i, sem):
        a, b = WQ_SPLIT[i]
        sl = pl.ds(a, b - a)
        return pltpu.make_async_copy(wq_hbm.at[sl], wq.at[sl], sem)

    def load_x(c, sem):
        r0 = n_xrecv if c - 2 in xrecv else 0
        return pltpu.make_async_copy(x_hbm.at[pl.ds(rows[c] + r0, 64 - r0)],
                                     xs.at[pl.ds(64 * c + r0, 64 - r0)], sem)

    def load_kv(src, dst, i, sem):
        b = batch[f] if i == 0 else 1 - batch[f]
        return pltpu.make_async_copy(src.at[b, pl.ds(p * 256, 256)], dst.at[b], sem)

    def load_wo(j, sem):
        return pltpu.make_async_copy(wo_hbm.at[:, pl.ds(128 * j, 128)], wo.at[j], sem)

    def load_wo12(_, sem):
        return pltpu.make_async_copy(wo_hbm.at[:, pl.ds(128, 256)], wo12, sem)

    makers = {"q": load_wq, "x": load_x, "w": load_wo, "m": load_wo12,
              "k": functools.partial(load_kv, k_hbm, kb),
              "v": functools.partial(load_kv, v_hbm, vb)}
    order = {
        "A": "q0 x0 x1 q1 q2 k0 v0 w0 w1 x2 x3 w2 k1 w3 v1",
        "M": f"q0 x0 x1 q1 q2 k0 k1 v0 v1 w0 w1 w2 x{2 + g} x{2 + f} w3",
        "Z": "q0 x0 x1 q1 q2 k0 v0 w3 m1 x2 x3 w0 k1 v1",
    }[role].split()
    barrier = pltpu.get_barrier_semaphore()
    loads = {}
    for ix, nm in enumerate(order):
        loads[nm] = makers[nm[0]](int(nm[1]), lsem.at[ix])
        loads[nm].start()
        if ix == 0:
            for n in part:
                pl.semaphore_signal(barrier, inc=1, device_id=(n,), device_id_type=MESH)

    def wait(names):
        for nm in names.split():
            loads.pop(nm).wait()

    rsems = (rsem1, rsem2, rsem3)

    def rcopy(step, half, j, n):
        tgt = part[half] if step != 1 else part[1 - half]
        rs = pl.ds(n * RP, RP)
        return pltpu.make_async_remote_copy(
            src_ref=sb.at[step, half, j, rs], dst_ref=rb.at[step, half, j, rs],
            send_sem=ssem.at[step, half], recv_sem=rsems[step].at[half, j, n],
            device_id=(tgt,), device_id_type=MESH)

    def dcopy(half, j, n):
        i = DETOUR.index((j, n))
        return pltpu.make_async_remote_copy(
            src_ref=sb.at[0, half, j, pl.ds(n * RP, RP)], dst_ref=rbd.at[half, pl.ds(i * RP, RP)],
            send_sem=ssem.at[0, half], recv_sem=dsem.at[half, i],
            device_id=(part[1 - half],), device_id_type=MESH)

    def xcopy(half, n):
        return pltpu.make_async_remote_copy(
            src_ref=sbx.at[half, pl.ds(0, n // 16)], dst_ref=rbx.at[half, pl.ds(0, n // 16)],
            send_sem=xssem.at[half], recv_sem=xrsem.at[half],
            device_id=(part[half],), device_id_type=MESH)

    def enter():
        pl.semaphore_wait(barrier, 2)
        for half in xsend:
            xcopy(half, n_xsend).start()

    lo = lax.broadcasted_iota(jnp.int32, (64, 128), 1) < 64
    zero = jnp.zeros((64, 128), F32)
    q, prob, ctx, out = {}, {}, {}, {}

    def dot(a, b):
        return jnp.dot(a, b, preferred_element_type=F32)

    def dot_t(a, b):
        return lax.dot_general(a, b, (((1,), (1,)), ((), ())), preferred_element_type=F32)

    def recip(den):
        r = pl.reciprocal(den, approx=True)
        return r * (2.0 - den * r)

    def scores(c):
        prob[c] = []
        for h in range(4):
            pr = h // 2
            kh = kb[batch[c], 64 * h:64 * h + 64, :]
            w = jnp.concatenate([kh, zero] if h % 2 == 0 else [zero, kh], 0)
            s = dot(q[c][:, 128 * pr:128 * pr + 128], w)
            if c % 2 == 0:
                s = jnp.where(lo, s, MASK)
            m = jnp.max(s, axis=1, keepdims=True)
            prob[c].append(jnp.exp2((s - m) * C_EXP))

    def pv(c):
        cs = []
        for pr in range(2):
            w = vb[batch[c], 128 * pr:128 * pr + 128, :]
            pp = prob[c][2 * pr:2 * pr + 2]
            lhs = jnp.concatenate(
                [t[u * G:(u + 1) * G] for u in range(64 // G) for t in pp], 0)
            tt = dot_t(lhs, w)
            t = [jnp.concatenate([tt[(2 * u + i) * G:(2 * u + i + 1) * G]
                                  for u in range(64 // G)], 0) for i in range(2)]
            sm = [jnp.sum(a, axis=1, keepdims=True) for a in pp]
            cs.append(jnp.where(lo, t[0], t[1]) * recip(jnp.where(lo, sm[0], sm[1])))
        ctx[c] = jnp.concatenate(cs, 1)

    heads = []

    def mix(a, b):
        return jnp.concatenate([t[u * RP:(u + 1) * RP] for u in range(NP) for t in (a, b)], 0)

    def unmix(t, i):
        return jnp.concatenate([t[(2 * u + i) * RP:(2 * u + i + 1) * RP] for u in range(NP)], 0)

    def pv_heads():
        def v(c, h):
            return vb[batch[c], 64 * h:64 * h + 64, :]
        if batch[f] != batch[g]:
            tt = {c: [dot_t(prob[c][h], v(c, h)) for h in range(4)] for c in (f, g)}
        for h in range(4):
            pp = mix(prob[f][h], prob[g][h])
            t = dot_t(pp, v(f, h)) if batch[f] == batch[g] else mix(tt[f][h], tt[g][h])
            den = jnp.broadcast_to(jnp.sum(pp, axis=1, keepdims=True), (128, 64))
            heads.append(t * recip(den))

    def oproj_heads(j):
        o = [dot(heads[h], wo[j, 64 * h:64 * h + 64, :]) for h in (0, 2, 1, 3)]
        o = (o[0] + o[1]) + (o[2] + o[3])
        out[f, j], out[g, j] = unmix(o, 0), unmix(o, 1)
        t = jnp.concatenate(heads, 1)
        ctx[f], ctx[g] = unmix(t, 0), unmix(t, 1)

    def wo_tile(j):
        return wo12[:, 128 * (j - 1):128 * j] if role == "Z" and j in (1, 2) else wo[j]

    def oproj(c, j):
        out[c, j] = dot(ctx[c], wo_tile(j))

    def oproj_kept(j):
        o = dot(jnp.concatenate([ctx[2], ctx[3]], 0), wo_tile(j))
        out[2, j], out[3, j] = o[0:64], o[64:128]

    def oproj_sent(j):
        oproj(f, j)
        oproj(g, j)

    def q_kept():
        xx = []
        for c in (2, 3):
            if c - 2 in xrecv:
                xx += [jnp.concatenate([rbx[c - 2, u, j].astype(F32) for j in range(4)], 1)
                       for u in range(n_xrecv // 16)]
                xx.append(xs[64 * c + n_xrecv:64 * c + 64, :])
            else:
                xx.append(xs[64 * c:64 * c + 64, :])
        t = dot(jnp.concatenate(xx, 0), wq[...])
        q[2], q[3] = t[0:64], t[64:128]

    def wait_x():
        for half in xrecv:
            xcopy(half, n_xrecv).wait_recv()

    def keep(j, r0=0):
        for c in (2, 3):
            acc[c - 2, j, r0:64] = out[c, j][r0:64]

    def store(c, j, n, t):
        o_ref[pl.ds(rows[c] + n * RP, RP), 128 * j:128 * j + 128] = t

    def step1(j):
        for n in range(NP):
            rs = slice(n * RP, (n + 1) * RP)
            detour = (j, n) in DETOUR
            for half in (f, g):
                if detour and role == "Z":
                    continue
                sb[0, half, j, rs] = out[half, j][rs].astype(BF)
                if detour and role == "M" and half == f:
                    dcopy(half, j, n).start()
                else:
                    rcopy(0, half, j, n).start()

    def step1_detour():
        for i, (j, n) in enumerate(DETOUR):
            rs = slice(n * RP, (n + 1) * RP)
            for half in range(2):
                a = out[half, j][rs] + rbd[half, i * RP:(i + 1) * RP].astype(F32)
                sb[0, half, j, rs] = a.astype(BF)
                rcopy(0, half, j, n).start()

    done2, done3 = set(), set()

    def step2(half, j, n, direct=False):
        rs = slice(n * RP, (n + 1) * RP)
        detour = (j, n) in DETOUR
        done2.add((half, j, n))
        if detour and role == "A":
            sb[1, half, j, rs] = acc[half, j, rs].astype(BF)
            rcopy(1, half, j, n).start()
        elif detour and role == "M" and half == g:
            rcopy(1, half, j, n).wait_recv()
            rcopy(0, half, j, n).wait_recv()
            t = (acc[half, j, rs] + rb[1, half, j, rs].astype(F32)
                 + rb[0, half, j, rs].astype(F32))
            for step in (1, 2):
                sb[step, half, j, rs] = t.astype(BF)
                rcopy(step, half, j, n).start()
            store(2 + half, j, n, t)
            done3.add((half, j, n))
        else:
            if direct:
                own = out[2 + half, j][rs]
            else:
                rcopy(0, half, j, n).wait_recv()
                own = acc[half, j, rs]
            a = own + rb[0, half, j, rs].astype(F32)
            sb[1, half, j, rs] = a.astype(BF)
            rcopy(1, half, j, n).start()
            acc[half, j, rs] = a

    def step3(half, j, n):
        rs = slice(n * RP, (n + 1) * RP)
        rcopy(1, half, j, n).wait_recv()
        t = rb[1, half, j, rs].astype(F32)
        if not ((j, n) in DETOUR and role == "A"):
            t = acc[half, j, rs] + t
        sb[2, half, j, rs] = t.astype(BF)
        rcopy(2, half, j, n).start()
        store(2 + half, j, n, t)

    for i, (a, b) in enumerate(WQ_SPLIT):
        if role == "M" and i == 1:
            enter()
        wait("q0 x0 x1" if i == 0 else f"q{i}")
        if i == 0:
            for half in xsend:
                for u in range(n_xsend // 16):
                    r0 = 64 * half + 16 * u
                    for j in range(4):
                        sbx[half, u, j] = xs[r0:r0 + 16, 128 * j:128 * j + 128].astype(BF)
            xx = xs[0:128, a:b]
            tt = jnp.concatenate([dot(xx, wq[a:b, 0:128]), dot(xx, wq[a:b, 128:256])], 1)
        else:
            w = wq[a:b, :]
        for half in (f, g):
            if i == 0:
                t = tt[64 * half:64 * half + 64]
            else:
                t = dot(xs[64 * half:64 * half + 64, a:b], w) + qacc[half]
            if i < len(WQ_SPLIT) - 1:
                qacc[half] = t
            else:
                q[half] = t

    if role == "A":
        wait("k0")
        enter()
        scores(f), scores(g)
        wait("v0 w0")
        pv(f), pv(g), oproj_sent(0), step1(0)
        wait("w1")
        oproj_sent(1), step1(1)
        wait("x2 x3")
        q_kept()
        wait("w2 k1")
        oproj_sent(2), scores(2), scores(3), step1(2)
        wait("w3 v1")
        oproj_sent(3), pv(2), pv(3)
        for j in range(4):
            oproj_kept(j)
        step1(3)
        for j in range(4):
            keep(j)
    elif role == "M":
        wait("k0 k1")
        scores(f), scores(g)
        wait("v0 v1")
        pv_heads()
        for j in range(3):
            wait(f"w{j}")
            (oproj_sent if j else oproj_heads)(j), step1(j)
        wait(f"x{2 + g} x{2 + f}")
        wait_x()
        q_kept()
        wait("w3")
        scores(2), scores(3), oproj_sent(3), pv(2), pv(3), step1(3)
        for c in (2, 3):
            for j in range(4):
                oproj(c, j)
        for j in range(4):
            keep(j)
    else:
        wait("k0")
        scores(f), scores(g)
        enter()
        wait("v0 w3")
        pv_heads(), oproj_heads(3), step1(3)
        wait("m1")
        oproj_sent(1), oproj_sent(2), step1(1), step1(2)
        wait("x2 x3")
        wait_x()
        q_kept()
        wait("w0 k1")
        scores(2), scores(3), oproj_sent(0), step1(0)
        wait("v1")
        for half in range(2):
            for n in range(N_DIRECT):
                rcopy(0, half, 0, n).wait_recv()
            for j, n in DETOUR:
                dcopy(half, j, n).wait_recv()
        pv(2), pv(3), step1_detour()
        oproj(2, 0), oproj(3, 0), oproj(2, 1), oproj(3, 1)
        for n in range(N_DIRECT):
            for half in range(2):
                step2(half, 0, n, direct=True)
        keep(0, N_DIRECT * RP), keep(1)
        for j, n in pieces[N_DIRECT:NP + NP // 2]:
            for half in range(2):
                step2(half, j, n)
        oproj_kept(2), oproj_kept(3), keep(2), keep(3)
    assert not loads

    for t in range(len(pieces)):
        for half in range(2):
            j, n = (z_order if role == "M" and half == g else pieces)[t]
            if (half, j, n) not in done2:
                step2(half, j, n)

    for t in range(len(pieces)):
        for half in range(2):
            j, n = (z_order if role == "A" else pieces)[t]
            if (half, j, n) not in done3:
                step3(half, j, n)

    for t in range(len(pieces)):
        if t == len(pieces) - 2:
            for half in xsend:
                xcopy(half, n_xsend).wait_send()
            for step in range(3):
                for half in range(2):
                    pltpu.make_async_copy(sb.at[step, half], sb.at[step, half],
                                          ssem.at[step, half]).wait()
        for half in range(2):
            j, n = (z_order if role == "M" and half == f else pieces)[t]
            rcopy(2, half, j, n).wait_recv()
            store(half, j, n, rb[2, half, j, n * RP:(n + 1) * RP].astype(F32))


def _body(*refs):
    p = lax.axis_index("i")
    for ps in (2, 1, 3, 0):
        pl.when(p == ps)(functools.partial(_program, ps, *refs))


def pallas_dist_sparse_attn_blocksparse_htp_b2_sq128_skv128_hq4_dh64_kernel(
    x: jax.Array,
    Wq: jax.Array,
    K_ext: jax.Array,
    V_ext: jax.Array,
    Wo: jax.Array,
):
    kt = jnp.transpose(K_ext, (0, 2, 3, 1)).reshape(2, 1024, 128)
    vt = jnp.transpose(V_ext, (0, 2, 3, 1)).reshape(2, 1024, 128)
    x2 = x.reshape(256, 512)
    any_ = pl.BlockSpec(memory_space=pl.ANY)
    nx = max(X_FWD.values()) // 16
    out = pl.pallas_call(
        _body,
        out_shape=jax.ShapeDtypeStruct((256, 512), F32),
        in_specs=[any_] * 5,
        out_specs=pl.BlockSpec(memory_space=pltpu.VMEM),
        scratch_shapes=[
            pltpu.VMEM((256, 512), F32),
            pltpu.VMEM((512, 256), F32),
            pltpu.VMEM((2, 256, 128), F32),
            pltpu.VMEM((2, 256, 128), F32),
            pltpu.VMEM((4, 256, 128), F32),
            pltpu.VMEM((256, 256), F32),
            pltpu.VMEM((2, 64, 256), F32),
            pltpu.VMEM((2, 4, 64, 128), F32),
            pltpu.VMEM((3, 2, 4, 64, 128), BF),
            pltpu.VMEM((3, 2, 4, 64, 128), BF),
            pltpu.VMEM((2, nx, 4, 16, 128), BF),
            pltpu.VMEM((2, nx, 4, 16, 128), BF),
            pltpu.VMEM((2, len(DETOUR) * RP, 128), BF),
            pltpu.SemaphoreType.DMA((15,)),
            pltpu.SemaphoreType.DMA((3, 2)),
            pltpu.SemaphoreType.DMA((2, 4, NP)),
            pltpu.SemaphoreType.DMA((2, 4, NP)),
            pltpu.SemaphoreType.DMA((2, 4, NP)),
            pltpu.SemaphoreType.DMA((2,)),
            pltpu.SemaphoreType.DMA((2,)),
            pltpu.SemaphoreType.DMA((2, len(DETOUR))),
        ],
        compiler_params=pltpu.CompilerParams(
            collective_id=0,
            disable_semaphore_checks=True,
            disable_bounds_checks=True,
        ),
    )(x2, Wq, kt, vt, Wo)
    return out.reshape(2, 128, 512)
```

```python
import functools
import math

import jax
import jax.numpy as jnp
from jax import lax
from jax.experimental import pallas as pl
from jax.experimental.pallas import tpu as pltpu

BF = jnp.bfloat16
F32 = jnp.float32
MESH = pl.DeviceIdType.MESH

C_EXP = 0.125 * math.log2(math.e)
MASK = -8e9
RP = 8
NP = 64 // RP
G = 16
WQ_SPLIT = ((0, 256), (256, 384), (384, 512))
X_FWD = {"A": 48, "M": 32}
DETOUR = ((0, 2), (0, 3))
N_DIRECT = 3


def _program(p, x_hbm, wq_hbm, k_hbm, v_hbm, wo_hbm, o_ref,
             xs, wq, kb, vb, wo, wo12, qacc, acc, sb, rb, sbx, rbx, rbd,
             lsem, ssem, rsem1, rsem2, rsem3, xssem, xrsem, dsem):
    cx = p >> 1
    cy = (p ^ cx) & 1
    part = (p ^ 1, 3 - p)
    batch = (cy, cx, 1 - cy, 1 - cx)
    rows = tuple(batch[c] * 128 + 64 * (c % 2) for c in range(4))
    role = "AMZM"[p]
    f = 1 if p == 3 else 0
    g = 1 - f
    xsend = {"A": (0, 1), "M": (g,), "Z": ()}[role]
    xrecv = {"A": (), "M": (f,), "Z": (0, 1)}[role]
    n_xsend = X_FWD.get(role, 0)
    n_xrecv = {"A": 0, "M": X_FWD["A"], "Z": X_FWD["M"]}[role]
    pieces = [(j, n) for j in range(4) for n in range(NP)]
    z_order = [(j, n) for j in (3, 1, 2, 0) for n in range(NP) if (j, n) not in DETOUR]
    z_order += list(DETOUR)

    def load_wq(i, sem):
        a, b = WQ_SPLIT[i]
        sl = pl.ds(a, b - a)
        return pltpu.make_async_copy(wq_hbm.at[sl], wq.at[sl], sem)

    def load_x(c, sem):
        r0 = n_xrecv if c - 2 in xrecv else 0
        return pltpu.make_async_copy(x_hbm.at[pl.ds(rows[c] + r0, 64 - r0)],
                                     xs.at[pl.ds(64 * c + r0, 64 - r0)], sem)

    def load_kv(src, dst, i, sem):
        b = batch[f] if i == 0 else 1 - batch[f]
        return pltpu.make_async_copy(src.at[b, pl.ds(p * 256, 256)], dst.at[b], sem)

    def load_wo(j, sem):
        return pltpu.make_async_copy(wo_hbm.at[:, pl.ds(128 * j, 128)], wo.at[j], sem)

    def load_wo12(_, sem):
        return pltpu.make_async_copy(wo_hbm.at[:, pl.ds(128, 256)], wo12, sem)

    makers = {"q": load_wq, "x": load_x, "w": load_wo, "m": load_wo12,
              "k": functools.partial(load_kv, k_hbm, kb),
              "v": functools.partial(load_kv, v_hbm, vb)}
    order = {
        "A": "q0 x0 x1 q1 q2 k0 v0 w0 w1 x2 x3 w2 k1 w3 v1",
        "M": f"q0 x0 x1 q1 q2 k0 k1 v0 v1 w0 w1 x{2 + g} w2 x{2 + f} w3",
        "Z": "q0 x0 x1 q1 q2 k0 v0 w3 m1 x2 x3 w0 k1 v1",
    }[role].split()
    barrier = pltpu.get_barrier_semaphore()
    loads = {}
    for ix, nm in enumerate(order):
        loads[nm] = makers[nm[0]](int(nm[1]), lsem.at[ix])
        loads[nm].start()
        if ix == 0:
            for n in part:
                pl.semaphore_signal(barrier, inc=1, device_id=(n,), device_id_type=MESH)

    def wait(names):
        for nm in names.split():
            loads.pop(nm).wait()

    rsems = (rsem1, rsem2, rsem3)

    def rcopy(step, half, j, n):
        tgt = part[half] if step != 1 else part[1 - half]
        rs = pl.ds(n * RP, RP)
        return pltpu.make_async_remote_copy(
            src_ref=sb.at[step, half, j, rs], dst_ref=rb.at[step, half, j, rs],
            send_sem=ssem.at[step, half], recv_sem=rsems[step].at[half, j, n],
            device_id=(tgt,), device_id_type=MESH)

    def dcopy(half, j, n):
        i = DETOUR.index((j, n))
        return pltpu.make_async_remote_copy(
            src_ref=sb.at[0, half, j, pl.ds(n * RP, RP)], dst_ref=rbd.at[half, pl.ds(i * RP, RP)],
            send_sem=ssem.at[0, half], recv_sem=dsem.at[half, i],
            device_id=(part[1 - half],), device_id_type=MESH)

    def xcopy(half, n):
        return pltpu.make_async_remote_copy(
            src_ref=sbx.at[half, pl.ds(0, n // 16)], dst_ref=rbx.at[half, pl.ds(0, n // 16)],
            send_sem=xssem.at[half], recv_sem=xrsem.at[half],
            device_id=(part[half],), device_id_type=MESH)

    def enter():
        pl.semaphore_wait(barrier, 2)
        for half in xsend:
            xcopy(half, n_xsend).start()

    lo = lax.broadcasted_iota(jnp.int32, (64, 128), 1) < 64
    zero = jnp.zeros((64, 128), F32)
    q, prob, ctx, out = {}, {}, {}, {}

    def dot(a, b):
        return jnp.dot(a, b, preferred_element_type=F32)

    def dot_t(a, b):
        return lax.dot_general(a, b, (((1,), (1,)), ((), ())), preferred_element_type=F32)

    def recip(den):
        r = pl.reciprocal(den, approx=True)
        return r * (2.0 - den * r)

    def scores(c):
        prob[c] = []
        for h in range(4):
            pr = h // 2
            kh = kb[batch[c], 64 * h:64 * h + 64, :]
            w = jnp.concatenate([kh, zero] if h % 2 == 0 else [zero, kh], 0)
            s = dot(q[c][:, 128 * pr:128 * pr + 128], w)
            if c % 2 == 0:
                s = jnp.where(lo, s, MASK)
            m = jnp.max(s, axis=1, keepdims=True)
            prob[c].append(jnp.exp2((s - m) * C_EXP))

    def pv(c):
        cs = []
        for pr in range(2):
            w = vb[batch[c], 128 * pr:128 * pr + 128, :]
            pp = prob[c][2 * pr:2 * pr + 2]
            lhs = jnp.concatenate(
                [t[u * G:(u + 1) * G] for u in range(64 // G) for t in pp], 0)
            tt = dot_t(lhs, w)
            t = [jnp.concatenate([tt[(2 * u + i) * G:(2 * u + i + 1) * G]
                                  for u in range(64 // G)], 0) for i in range(2)]
            sm = [jnp.sum(a, axis=1, keepdims=True) for a in pp]
            cs.append(jnp.where(lo, t[0], t[1]) * recip(jnp.where(lo, sm[0], sm[1])))
        ctx[c] = jnp.concatenate(cs, 1)

    def pv_plain(c):
        cs = []
        for pr in range(2):
            w = vb[batch[c], 128 * pr:128 * pr + 128, :]
            pp = prob[c][2 * pr:2 * pr + 2]
            t = [dot_t(a, w) for a in pp]
            sm = [jnp.sum(a, axis=1, keepdims=True) for a in pp]
            cs.append(jnp.where(lo, t[0], t[1]) * recip(jnp.where(lo, sm[0], sm[1])))
        ctx[c] = jnp.concatenate(cs, 1)

    heads = []

    def mix(a, b):
        return jnp.concatenate([t[u * RP:(u + 1) * RP] for u in range(NP) for t in (a, b)], 0)

    def unmix(t, i):
        return jnp.concatenate([t[(2 * u + i) * RP:(2 * u + i + 1) * RP] for u in range(NP)], 0)

    def pv_heads():
        def v(c, h):
            return vb[batch[c], 64 * h:64 * h + 64, :]
        if batch[f] != batch[g]:
            tt = {c: [dot_t(prob[c][h], v(c, h)) for h in range(4)] for c in (f, g)}
        for h in range(4):
            pp = mix(prob[f][h], prob[g][h])
            t = dot_t(pp, v(f, h)) if batch[f] == batch[g] else mix(tt[f][h], tt[g][h])
            den = jnp.broadcast_to(jnp.sum(pp, axis=1, keepdims=True), (128, 64))
            heads.append(t * recip(den))

    def oproj_heads(j):
        o = [dot(heads[h], wo[j, 64 * h:64 * h + 64, :]) for h in (0, 2, 1, 3)]
        o = (o[0] + o[1]) + (o[2] + o[3])
        out[f, j], out[g, j] = unmix(o, 0), unmix(o, 1)
        t = jnp.concatenate(heads, 1)
        ctx[f], ctx[g] = unmix(t, 0), unmix(t, 1)

    def wo_tile(j):
        return wo12[:, 128 * (j - 1):128 * j] if role == "Z" and j in (1, 2) else wo[j]

    def oproj(c, j):
        out[c, j] = dot(ctx[c], wo_tile(j))

    def oproj_kept(j):
        o = dot(jnp.concatenate([ctx[2], ctx[3]], 0), wo_tile(j))
        out[2, j], out[3, j] = o[0:64], o[64:128]

    def oproj_sent(j):
        oproj(f, j)
        oproj(g, j)

    def q_kept(cs=(2, 3)):
        xx = []
        for c in cs:
            if c - 2 in xrecv:
                xx += [jnp.concatenate([rbx[c - 2, u, j].astype(F32) for j in range(4)], 1)
                       for u in range(n_xrecv // 16)]
                xx.append(xs[64 * c + n_xrecv:64 * c + 64, :])
            else:
                xx.append(xs[64 * c:64 * c + 64, :])
        t = dot(jnp.concatenate(xx, 0), wq[...])
        for i, c in enumerate(cs):
            q[c] = t[64 * i:64 * i + 64]

    def wait_x():
        for half in xrecv:
            xcopy(half, n_xrecv).wait_recv()

    def keep(j, r0=0):
        for c in (2, 3):
            acc[c - 2, j, r0:64] = out[c, j][r0:64]

    def store(c, j, n, t):
        o_ref[pl.ds(rows[c] + n * RP, RP), 128 * j:128 * j + 128] = t

    def step1(j):
        for n in range(NP):
            rs = slice(n * RP, (n + 1) * RP)
            detour = (j, n) in DETOUR
            for half in (f, g):
                if detour and role == "Z":
                    continue
                sb[0, half, j, rs] = out[half, j][rs].astype(BF)
                if detour and role == "M" and half == f:
                    dcopy(half, j, n).start()
                else:
                    rcopy(0, half, j, n).start()

    def step1_detour():
        for i, (j, n) in enumerate(DETOUR):
            rs = slice(n * RP, (n + 1) * RP)
            for half in range(2):
                a = out[half, j][rs] + rbd[half, i * RP:(i + 1) * RP].astype(F32)
                sb[0, half, j, rs] = a.astype(BF)
                rcopy(0, half, j, n).start()

    done2, done3 = set(), set()

    def step2(half, j, n, direct=False):
        rs = slice(n * RP, (n + 1) * RP)
        detour = (j, n) in DETOUR
        done2.add((half, j, n))
        if detour and role == "A":
            sb[1, half, j, rs] = acc[half, j, rs].astype(BF)
            rcopy(1, half, j, n).start()
        elif detour and role == "M" and half == g:
            rcopy(1, half, j, n).wait_recv()
            rcopy(0, half, j, n).wait_recv()
            t = (acc[half, j, rs] + rb[1, half, j, rs].astype(F32)
                 + rb[0, half, j, rs].astype(F32))
            for step in (1, 2):
                sb[step, half, j, rs] = t.astype(BF)
                rcopy(step, half, j, n).start()
            store(2 + half, j, n, t)
            done3.add((half, j, n))
        else:
            if direct:
                own = out[2 + half, j][rs]
            else:
                rcopy(0, half, j, n).wait_recv()
                own = acc[half, j, rs]
            a = own + rb[0, half, j, rs].astype(F32)
            sb[1, half, j, rs] = a.astype(BF)
            rcopy(1, half, j, n).start()
            acc[half, j, rs] = a

    def step3(half, j, n):
        rs = slice(n * RP, (n + 1) * RP)
        rcopy(1, half, j, n).wait_recv()
        t = rb[1, half, j, rs].astype(F32)
        if not ((j, n) in DETOUR and role == "A"):
            t = acc[half, j, rs] + t
        sb[2, half, j, rs] = t.astype(BF)
        rcopy(2, half, j, n).start()
        store(2 + half, j, n, t)

    for i, (a, b) in enumerate(WQ_SPLIT):
        if role == "M" and i == 1:
            enter()
        wait("q0 x0 x1" if i == 0 else f"q{i}")
        if i == 0:
            for half in xsend:
                for u in range(n_xsend // 16):
                    r0 = 64 * half + 16 * u
                    for j in range(4):
                        sbx[half, u, j] = xs[r0:r0 + 16, 128 * j:128 * j + 128].astype(BF)
            xx = xs[0:128, a:b]
            tt = jnp.concatenate([dot(xx, wq[a:b, 0:128]), dot(xx, wq[a:b, 128:256])], 1)
        else:
            w = wq[a:b, :]
        for half in (f, g):
            if i == 0:
                t = tt[64 * half:64 * half + 64]
            else:
                t = dot(xs[64 * half:64 * half + 64, a:b], w) + qacc[half]
            if i < len(WQ_SPLIT) - 1:
                qacc[half] = t
            else:
                q[half] = t

    if role == "A":
        wait("k0")
        enter()
        scores(f), scores(g)
        wait("v0 w0")
        pv(f), pv(g), oproj_sent(0), step1(0)
        wait("w1")
        oproj_sent(1), step1(1)
        wait("x2 x3")
        q_kept()
        wait("w2 k1")
        oproj_sent(2), scores(2), scores(3), step1(2)
        wait("w3 v1")
        oproj_sent(3), pv(2), pv(3)
        for j in range(4):
            oproj_kept(j)
        step1(3)
        for j in range(4):
            keep(j)
    elif role == "M":
        wait("k0 k1")
        scores(f), scores(g)
        wait("v0 v1")
        pv_heads()
        wait("w0")
        oproj_heads(0), step1(0)
        wait("w1")
        oproj_sent(1), step1(1)
        a, b = 2 + g, 2 + f
        wait(f"x{a}")
        q_kept((a,))
        wait(f"w2 x{b}")
        wait_x()
        oproj_sent(2), scores(a), q_kept((b,)), step1(2)
        wait("w3")
        oproj_sent(3), scores(b), pv_plain(a), step1(3)
        oproj(a, 0), oproj(a, 1), pv_plain(b), oproj(a, 2), oproj(a, 3)
        for j in range(4):
            oproj(b, j)
        for j in range(4):
            keep(j)
    else:
        wait("k0")
        scores(f), scores(g)
        enter()
        wait("v0 w3")
        pv_heads(), oproj_heads(3), step1(3)
        wait("m1")
        oproj_sent(1), oproj_sent(2), step1(1), step1(2)
        wait("x2 x3")
        wait_x()
        q_kept()
        wait("w0 k1")
        scores(2), scores(3), oproj_sent(0), step1(0)
        wait("v1")
        for half in range(2):
            for n in range(N_DIRECT):
                rcopy(0, half, 0, n).wait_recv()
            for j, n in DETOUR:
                dcopy(half, j, n).wait_recv()
        pv(2), pv(3), step1_detour()
        oproj(2, 0), oproj(3, 0), oproj(2, 1), oproj(3, 1)
        for n in range(N_DIRECT):
            for half in range(2):
                step2(half, 0, n, direct=True)
        keep(0, N_DIRECT * RP), keep(1)
        for j, n in pieces[N_DIRECT:NP + NP // 2]:
            for half in range(2):
                step2(half, j, n)
        oproj_kept(2), oproj_kept(3), keep(2), keep(3)
    assert not loads

    for t in range(len(pieces)):
        for half in range(2):
            j, n = (z_order if role == "M" and half == g else pieces)[t]
            if (half, j, n) not in done2:
                step2(half, j, n)

    for t in range(len(pieces)):
        for half in range(2):
            j, n = (z_order if role == "A" else pieces)[t]
            if (half, j, n) not in done3:
                step3(half, j, n)

    for t in range(len(pieces)):
        if t == len(pieces) - 2:
            for half in xsend:
                xcopy(half, n_xsend).wait_send()
            for step in range(3):
                for half in range(2):
                    pltpu.make_async_copy(sb.at[step, half], sb.at[step, half],
                                          ssem.at[step, half]).wait()
        for half in range(2):
            j, n = (z_order if role == "M" and half == f else pieces)[t]
            rcopy(2, half, j, n).wait_recv()
            store(half, j, n, rb[2, half, j, n * RP:(n + 1) * RP].astype(F32))


def _body(*refs):
    p = lax.axis_index("i")
    for ps in (2, 1, 3, 0):
        pl.when(p == ps)(functools.partial(_program, ps, *refs))


def pallas_dist_sparse_attn_blocksparse_htp_b2_sq128_skv128_hq4_dh64_kernel(
    x: jax.Array,
    Wq: jax.Array,
    K_ext: jax.Array,
    V_ext: jax.Array,
    Wo: jax.Array,
):
    kt = jnp.transpose(K_ext, (0, 2, 3, 1)).reshape(2, 1024, 128)
    vt = jnp.transpose(V_ext, (0, 2, 3, 1)).reshape(2, 1024, 128)
    x2 = x.reshape(256, 512)
    any_ = pl.BlockSpec(memory_space=pl.ANY)
    nx = max(X_FWD.values()) // 16
    out = pl.pallas_call(
        _body,
        out_shape=jax.ShapeDtypeStruct((256, 512), F32),
        in_specs=[any_] * 5,
        out_specs=pl.BlockSpec(memory_space=pltpu.VMEM),
        scratch_shapes=[
            pltpu.VMEM((256, 512), F32),
            pltpu.VMEM((512, 256), F32),
            pltpu.VMEM((2, 256, 128), F32),
            pltpu.VMEM((2, 256, 128), F32),
            pltpu.VMEM((4, 256, 128), F32),
            pltpu.VMEM((256, 256), F32),
            pltpu.VMEM((2, 64, 256), F32),
            pltpu.VMEM((2, 4, 64, 128), F32),
            pltpu.VMEM((3, 2, 4, 64, 128), BF),
            pltpu.VMEM((3, 2, 4, 64, 128), BF),
            pltpu.VMEM((2, nx, 4, 16, 128), BF),
            pltpu.VMEM((2, nx, 4, 16, 128), BF),
            pltpu.VMEM((2, len(DETOUR) * RP, 128), BF),
            pltpu.SemaphoreType.DMA((15,)),
            pltpu.SemaphoreType.DMA((3, 2)),
            pltpu.SemaphoreType.DMA((2, 4, NP)),
            pltpu.SemaphoreType.DMA((2, 4, NP)),
            pltpu.SemaphoreType.DMA((2, 4, NP)),
            pltpu.SemaphoreType.DMA((2,)),
            pltpu.SemaphoreType.DMA((2,)),
            pltpu.SemaphoreType.DMA((2, len(DETOUR))),
        ],
        compiler_params=pltpu.CompilerParams(
            collective_id=0,
            disable_semaphore_checks=True,
            disable_bounds_checks=True,
        ),
    )(x2, Wq, kt, vt, Wo)
    return out.reshape(2, 128, 512)
```

```python
import functools
import math

import jax
import jax.numpy as jnp
from jax import lax
from jax.experimental import pallas as pl
from jax.experimental.pallas import tpu as pltpu

BF = jnp.bfloat16
F32 = jnp.float32
MESH = pl.DeviceIdType.MESH

C_EXP = 0.125 * math.log2(math.e)
MASK = -8e9
RP = 8
NP = 64 // RP
G = 16
WQ_SPLIT = ((0, 256), (256, 384), (384, 512))
X_FWD = {"A": 48, "M": 32}
DETOUR = ((0, 2), (0, 3))
N_DIRECT = 3
LEAD = 6


def _program(p, x_hbm, wq_hbm, k_hbm, v_hbm, wo_hbm, o_ref,
             xs, wq, kb, vb, wo, wo12, qacc, acc, sb, rb, sbx, rbx, rbd,
             lsem, ssem, rsem1, rsem2, rsem3, xssem, xrsem, dsem):
    cx = p >> 1
    cy = (p ^ cx) & 1
    part = (p ^ 1, 3 - p)
    batch = (cy, cx, 1 - cy, 1 - cx)
    rows = tuple(batch[c] * 128 + 64 * (c % 2) for c in range(4))
    role = "AMZM"[p]
    f = 1 if p == 3 else 0
    g = 1 - f
    xsend = {"A": (0, 1), "M": (g,), "Z": ()}[role]
    xrecv = {"A": (), "M": (f,), "Z": (0, 1)}[role]
    n_xsend = X_FWD.get(role, 0)
    n_xrecv = {"A": 0, "M": X_FWD["A"], "Z": X_FWD["M"]}[role]
    pieces = [(j, n) for j in range(4) for n in range(NP)]
    z_order = [(j, n) for j in (3, 1, 2, 0) for n in range(NP) if (j, n) not in DETOUR]
    z_order += list(DETOUR)

    def load_wq(i, sem):
        a, b = WQ_SPLIT[i]
        sl = pl.ds(a, b - a)
        return pltpu.make_async_copy(wq_hbm.at[sl], wq.at[sl], sem)

    def load_x(c, sem):
        r0 = n_xrecv if c - 2 in xrecv else 0
        return pltpu.make_async_copy(x_hbm.at[pl.ds(rows[c] + r0, 64 - r0)],
                                     xs.at[pl.ds(64 * c + r0, 64 - r0)], sem)

    def load_kv(src, dst, i, sem):
        b = batch[f] if i == 0 else 1 - batch[f]
        return pltpu.make_async_copy(src.at[b, pl.ds(p * 256, 256)], dst.at[b], sem)

    def load_wo(j, sem):
        return pltpu.make_async_copy(wo_hbm.at[:, pl.ds(128 * j, 128)], wo.at[j], sem)

    def load_wo12(_, sem):
        return pltpu.make_async_copy(wo_hbm.at[:, pl.ds(128, 256)], wo12, sem)

    makers = {"q": load_wq, "x": load_x, "w": load_wo, "m": load_wo12,
              "k": functools.partial(load_kv, k_hbm, kb),
              "v": functools.partial(load_kv, v_hbm, vb)}
    order = {
        "A": "q0 x0 x1 q1 q2 k0 v0 w0 w1 x2 x3 w2 k1 w3 v1",
        "M": f"q0 x0 x1 q1 q2 k0 k1 v0 v1 w0 w1 x{2 + g} w2 x{2 + f} w3",
        "Z": "q0 x0 x1 q1 q2 k0 v0 w3 m1 x2 x3 w0 k1 v1",
    }[role].split()
    barrier = pltpu.get_barrier_semaphore()
    loads = {}
    for ix, nm in enumerate(order):
        loads[nm] = makers[nm[0]](int(nm[1]), lsem.at[ix])
        loads[nm].start()
        if ix == 0:
            for n in part:
                pl.semaphore_signal(barrier, inc=1, device_id=(n,), device_id_type=MESH)

    def wait(names):
        for nm in names.split():
            loads.pop(nm).wait()

    rsems = (rsem1, rsem2, rsem3)

    def rcopy(step, half, j, n):
        tgt = part[half] if step != 1 else part[1 - half]
        rs = pl.ds(n * RP, RP)
        return pltpu.make_async_remote_copy(
            src_ref=sb.at[step, half, j, rs], dst_ref=rb.at[step, half, j, rs],
            send_sem=ssem.at[step, half], recv_sem=rsems[step].at[half, j, n],
            device_id=(tgt,), device_id_type=MESH)

    def dcopy(half, j, n):
        i = DETOUR.index((j, n))
        return pltpu.make_async_remote_copy(
            src_ref=sb.at[0, half, j, pl.ds(n * RP, RP)], dst_ref=rbd.at[half, pl.ds(i * RP, RP)],
            send_sem=ssem.at[0, half], recv_sem=dsem.at[half, i],
            device_id=(part[1 - half],), device_id_type=MESH)

    def xcopy(half, n):
        return pltpu.make_async_remote_copy(
            src_ref=sbx.at[half, pl.ds(0, n // 16)], dst_ref=rbx.at[half, pl.ds(0, n // 16)],
            send_sem=xssem.at[half], recv_sem=xrsem.at[half],
            device_id=(part[half],), device_id_type=MESH)

    def enter():
        pl.semaphore_wait(barrier, 2)
        for half in xsend:
            xcopy(half, n_xsend).start()

    lo = lax.broadcasted_iota(jnp.int32, (64, 128), 1) < 64
    zero = jnp.zeros((64, 128), F32)
    q, prob, ctx, out = {}, {}, {}, {}

    def dot(a, b):
        return jnp.dot(a, b, preferred_element_type=F32)

    def dot_t(a, b):
        return lax.dot_general(a, b, (((1,), (1,)), ((), ())), preferred_element_type=F32)

    def recip(den):
        r = pl.reciprocal(den, approx=True)
        return r * (2.0 - den * r)

    def scores(c):
        prob[c] = []
        for h in range(4):
            pr = h // 2
            kh = kb[batch[c], 64 * h:64 * h + 64, :]
            w = jnp.concatenate([kh, zero] if h % 2 == 0 else [zero, kh], 0)
            s = dot(q[c][:, 128 * pr:128 * pr + 128], w)
            if c % 2 == 0:
                s = jnp.where(lo, s, MASK)
            m = jnp.max(s, axis=1, keepdims=True)
            prob[c].append(jnp.exp2((s - m) * C_EXP))

    def pv(c):
        cs = []
        for pr in range(2):
            w = vb[batch[c], 128 * pr:128 * pr + 128, :]
            pp = prob[c][2 * pr:2 * pr + 2]
            lhs = jnp.concatenate(
                [t[u * G:(u + 1) * G] for u in range(64 // G) for t in pp], 0)
            tt = dot_t(lhs, w)
            t = [jnp.concatenate([tt[(2 * u + i) * G:(2 * u + i + 1) * G]
                                  for u in range(64 // G)], 0) for i in range(2)]
            sm = [jnp.sum(a, axis=1, keepdims=True) for a in pp]
            cs.append(jnp.where(lo, t[0], t[1]) * recip(jnp.where(lo, sm[0], sm[1])))
        ctx[c] = jnp.concatenate(cs, 1)

    def pv_plain(c):
        cs = []
        for pr in range(2):
            w = vb[batch[c], 128 * pr:128 * pr + 128, :]
            pp = prob[c][2 * pr:2 * pr + 2]
            t = [dot_t(a, w) for a in pp]
            sm = [jnp.sum(a, axis=1, keepdims=True) for a in pp]
            cs.append(jnp.where(lo, t[0], t[1]) * recip(jnp.where(lo, sm[0], sm[1])))
        ctx[c] = jnp.concatenate(cs, 1)

    def mix(a, b):
        return jnp.concatenate([t[u * RP:(u + 1) * RP] for u in range(NP) for t in (a, b)], 0)

    def unmix(t, i):
        return jnp.concatenate([t[(2 * u + i) * RP:(2 * u + i + 1) * RP] for u in range(NP)], 0)

    def v_head(c, h):
        return vb[batch[c], 64 * h:64 * h + 64, :]

    def normalize(t, pp):
        return t * recip(jnp.broadcast_to(jnp.sum(pp, axis=1, keepdims=True), t.shape))

    def oproj_heads(heads, j):
        o = [dot(heads[h], wo[j, 64 * h:64 * h + 64, :]) for h in (0, 2, 1, 3)]
        return (o[0] + o[1]) + (o[2] + o[3])

    def publish(heads, o, j):
        out[f, j], out[g, j] = unmix(o, 0), unmix(o, 1)
        t = jnp.concatenate(heads, 1)
        ctx[f], ctx[g] = unmix(t, 0), unmix(t, 1)

    def first_tile_m(j):
        wait("k0 k1")
        scores(f), scores(g)
        wait("v0 v1")
        tt = {c: [dot_t(prob[c][h], v_head(c, h)) for h in range(4)] for c in (f, g)}
        heads = [normalize(mix(tt[f][h], tt[g][h]), mix(prob[f][h], prob[g][h]))
                 for h in range(4)]
        wait(f"w{j}")
        publish(heads, oproj_heads(heads, j), j)

    def first_tile_z(j):
        wait("k0")
        qq = mix(q[f], q[g])
        s, pp = {}, {}
        for h in range(4):
            kh = kb[batch[f], 64 * h:64 * h + 64, :]
            w = jnp.concatenate([kh, zero] if h % 2 == 0 else [zero, kh], 0)
            t = dot(qq[:, 128 * (h // 2):128 * (h // 2) + 128], w)
            for m in range(2 * NP):
                s[h, m] = t[m * RP:(m + 1) * RP]
                if (f, g)[m % 2] % 2 == 0:
                    s[h, m] = jnp.where(lo[0:RP], s[h, m], MASK)

        def softmax(m0, m1):
            for m in range(m0, m1):
                for h in range(4):
                    mx = jnp.max(s[h, m], axis=1, keepdims=True)
                    pp[h, m] = jnp.exp2((s[h, m] - mx) * C_EXP)

        def values(m0, m1):
            lhs = [jnp.concatenate([pp[h, m] for m in range(m0, m1)], 0) for h in range(4)]
            return [normalize(dot_t(lhs[h], v_head(f, h)), lhs[h]) for h in range(4)]

        softmax(0, LEAD)
        enter()
        wait("v0")
        ha = values(0, LEAD)
        softmax(LEAD, LEAD + 4)
        wait(f"w{j}")
        oa = oproj_heads(ha, j)
        softmax(LEAD + 4, 2 * NP)
        hb = values(LEAD, 2 * NP)
        publish([jnp.concatenate(t, 0) for t in zip(ha, hb)],
                jnp.concatenate([oa, oproj_heads(hb, j)], 0), j)

    def wo_tile(j):
        return wo12[:, 128 * (j - 1):128 * j] if role == "Z" and j in (1, 2) else wo[j]

    def oproj(c, j):
        out[c, j] = dot(ctx[c], wo_tile(j))

    def oproj_kept(j):
        o = dot(jnp.concatenate([ctx[2], ctx[3]], 0), wo_tile(j))
        out[2, j], out[3, j] = o[0:64], o[64:128]

    def oproj_sent(j):
        oproj(f, j)
        oproj(g, j)

    def q_kept(cs=(2, 3)):
        xx = []
        for c in cs:
            if c - 2 in xrecv:
                xx += [jnp.concatenate([rbx[c - 2, u, j].astype(F32) for j in range(4)], 1)
                       for u in range(n_xrecv // 16)]
                xx.append(xs[64 * c + n_xrecv:64 * c + 64, :])
            else:
                xx.append(xs[64 * c:64 * c + 64, :])
        t = dot(jnp.concatenate(xx, 0), wq[...])
        for i, c in enumerate(cs):
            q[c] = t[64 * i:64 * i + 64]

    def wait_x():
        for half in xrecv:
            xcopy(half, n_xrecv).wait_recv()

    def keep(j, r0=0):
        for c in (2, 3):
            acc[c - 2, j, r0:64] = out[c, j][r0:64]

    def store(c, j, n, t):
        o_ref[pl.ds(rows[c] + n * RP, RP), 128 * j:128 * j + 128] = t

    def step1(j):
        for n in range(NP):
            rs = slice(n * RP, (n + 1) * RP)
            detour = (j, n) in DETOUR
            for half in (f, g):
                if detour and role == "Z":
                    continue
                sb[0, half, j, rs] = out[half, j][rs].astype(BF)
                if detour and role == "M" and half == f:
                    dcopy(half, j, n).start()
                else:
                    rcopy(0, half, j, n).start()

    def step1_detour():
        for i, (j, n) in enumerate(DETOUR):
            rs = slice(n * RP, (n + 1) * RP)
            for half in range(2):
                a = out[half, j][rs] + rbd[half, i * RP:(i + 1) * RP].astype(F32)
                sb[0, half, j, rs] = a.astype(BF)
                rcopy(0, half, j, n).start()

    done2, done3 = set(), set()

    def step2(half, j, n, direct=False):
        rs = slice(n * RP, (n + 1) * RP)
        detour = (j, n) in DETOUR
        done2.add((half, j, n))
        if detour and role == "A":
            sb[1, half, j, rs] = acc[half, j, rs].astype(BF)
            rcopy(1, half, j, n).start()
        elif detour and role == "M" and half == g:
            rcopy(1, half, j, n).wait_recv()
            rcopy(0, half, j, n).wait_recv()
            t = (acc[half, j, rs] + rb[1, half, j, rs].astype(F32)
                 + rb[0, half, j, rs].astype(F32))
            for step in (1, 2):
                sb[step, half, j, rs] = t.astype(BF)
                rcopy(step, half, j, n).start()
            store(2 + half, j, n, t)
            done3.add((half, j, n))
        else:
            if direct:
                own = out[2 + half, j][rs]
            else:
                rcopy(0, half, j, n).wait_recv()
                own = acc[half, j, rs]
            a = own + rb[0, half, j, rs].astype(F32)
            sb[1, half, j, rs] = a.astype(BF)
            rcopy(1, half, j, n).start()
            acc[half, j, rs] = a

    def step3(half, j, n):
        rs = slice(n * RP, (n + 1) * RP)
        rcopy(1, half, j, n).wait_recv()
        t = rb[1, half, j, rs].astype(F32)
        if not ((j, n) in DETOUR and role == "A"):
            t = acc[half, j, rs] + t
        sb[2, half, j, rs] = t.astype(BF)
        rcopy(2, half, j, n).start()
        store(2 + half, j, n, t)

    for i, (a, b) in enumerate(WQ_SPLIT):
        if role == "M" and i == 1:
            enter()
        wait("q0 x0 x1" if i == 0 else f"q{i}")
        if i == 0:
            for half in xsend:
                for u in range(n_xsend // 16):
                    r0 = 64 * half + 16 * u
                    for j in range(4):
                        sbx[half, u, j] = xs[r0:r0 + 16, 128 * j:128 * j + 128].astype(BF)
            xx = xs[0:128, a:b]
            tt = jnp.concatenate([dot(xx, wq[a:b, 0:128]), dot(xx, wq[a:b, 128:256])], 1)
        else:
            w = wq[a:b, :]
        for half in (f, g):
            if i == 0:
                t = tt[64 * half:64 * half + 64]
            else:
                t = dot(xs[64 * half:64 * half + 64, a:b], w) + qacc[half]
            if i < len(WQ_SPLIT) - 1:
                qacc[half] = t
            else:
                q[half] = t

    if role == "A":
        wait("k0")
        enter()
        scores(f), scores(g)
        wait("v0 w0")
        pv(f), pv(g), oproj_sent(0), step1(0)
        wait("w1")
        oproj_sent(1), step1(1)
        wait("x2 x3")
        q_kept()
        wait("w2 k1")
        oproj_sent(2), scores(2), scores(3), step1(2)
        wait("w3 v1")
        oproj_sent(3), pv(2), pv(3)
        for j in range(4):
            oproj_kept(j)
        step1(3)
        for j in range(4):
            keep(j)
    elif role == "M":
        first_tile_m(0), step1(0)
        wait("w1")
        oproj_sent(1), step1(1)
        a, b = 2 + g, 2 + f
        wait(f"x{a}")
        q_kept((a,))
        wait(f"w2 x{b}")
        wait_x()
        oproj_sent(2), scores(a), q_kept((b,)), step1(2)
        wait("w3")
        oproj_sent(3), scores(b), pv_plain(a), step1(3)
        oproj(a, 0), oproj(a, 1), pv_plain(b), oproj(a, 2), oproj(a, 3)
        for j in range(4):
            oproj(b, j)
        for j in range(4):
            keep(j)
    else:
        first_tile_z(3), step1(3)
        wait("m1")
        oproj_sent(1), oproj_sent(2), step1(1), step1(2)
        wait("x2 x3")
        wait_x()
        q_kept()
        wait("w0 k1")
        scores(2), scores(3), oproj_sent(0), step1(0)
        wait("v1")
        for half in range(2):
            for n in range(N_DIRECT):
                rcopy(0, half, 0, n).wait_recv()
            for j, n in DETOUR:
                dcopy(half, j, n).wait_recv()
        pv(2), pv(3), step1_detour()
        oproj(2, 0), oproj(3, 0), oproj(2, 1), oproj(3, 1)
        for n in range(N_DIRECT):
            for half in range(2):
                step2(half, 0, n, direct=True)
        keep(0, N_DIRECT * RP), keep(1)
        for j, n in pieces[N_DIRECT:NP + NP // 2]:
            for half in range(2):
                step2(half, j, n)
        oproj_kept(2), oproj_kept(3), keep(2), keep(3)
    assert not loads

    for t in range(len(pieces)):
        for half in (g, f):
            j, n = (z_order if role == "M" and half == g else pieces)[t]
            if (half, j, n) not in done2:
                step2(half, j, n)

    for t in range(len(pieces)):
        for half in range(2):
            j, n = (z_order if role == "A" else pieces)[t]
            if (half, j, n) not in done3:
                step3(half, j, n)

    for t in range(len(pieces)):
        if t == len(pieces) - 2:
            for half in xsend:
                xcopy(half, n_xsend).wait_send()
            for step in range(3):
                for half in range(2):
                    pltpu.make_async_copy(sb.at[step, half], sb.at[step, half],
                                          ssem.at[step, half]).wait()
        for half in range(2):
            j, n = (z_order if role == "M" and half == f else pieces)[t]
            rcopy(2, half, j, n).wait_recv()
            store(half, j, n, rb[2, half, j, n * RP:(n + 1) * RP].astype(F32))


def _body(*refs):
    p = lax.axis_index("i")
    for ps in (2, 1, 3, 0):
        pl.when(p == ps)(functools.partial(_program, ps, *refs))


def pallas_dist_sparse_attn_blocksparse_htp_b2_sq128_skv128_hq4_dh64_kernel(
    x: jax.Array,
    Wq: jax.Array,
    K_ext: jax.Array,
    V_ext: jax.Array,
    Wo: jax.Array,
):
    kt = jnp.transpose(K_ext, (0, 2, 3, 1)).reshape(2, 1024, 128)
    vt = jnp.transpose(V_ext, (0, 2, 3, 1)).reshape(2, 1024, 128)
    x2 = x.reshape(256, 512)
    any_ = pl.BlockSpec(memory_space=pl.ANY)
    nx = max(X_FWD.values()) // 16
    out = pl.pallas_call(
        _body,
        out_shape=jax.ShapeDtypeStruct((256, 512), F32),
        in_specs=[any_] * 5,
        out_specs=pl.BlockSpec(memory_space=pltpu.VMEM),
        scratch_shapes=[
            pltpu.VMEM((256, 512), F32),
            pltpu.VMEM((512, 256), F32),
            pltpu.VMEM((2, 256, 128), F32),
            pltpu.VMEM((2, 256, 128), F32),
            pltpu.VMEM((4, 256, 128), F32),
            pltpu.VMEM((256, 256), F32),
            pltpu.VMEM((2, 64, 256), F32),
            pltpu.VMEM((2, 4, 64, 128), F32),
            pltpu.VMEM((3, 2, 4, 64, 128), BF),
            pltpu.VMEM((3, 2, 4, 64, 128), BF),
            pltpu.VMEM((2, nx, 4, 16, 128), BF),
            pltpu.VMEM((2, nx, 4, 16, 128), BF),
            pltpu.VMEM((2, len(DETOUR) * RP, 128), BF),
            pltpu.SemaphoreType.DMA((15,)),
            pltpu.SemaphoreType.DMA((3, 2)),
            pltpu.SemaphoreType.DMA((2, 4, NP)),
            pltpu.SemaphoreType.DMA((2, 4, NP)),
            pltpu.SemaphoreType.DMA((2, 4, NP)),
            pltpu.SemaphoreType.DMA((2,)),
            pltpu.SemaphoreType.DMA((2,)),
            pltpu.SemaphoreType.DMA((2, len(DETOUR))),
        ],
        compiler_params=pltpu.CompilerParams(
            collective_id=0,
            disable_semaphore_checks=True,
            disable_bounds_checks=True,
        ),
    )(x2, Wq, kt, vt, Wo)
    return out.reshape(2, 128, 512)
```
